```python
import numpy as np

kernel_name = "dist_ag_xy_y_m65536_n1024"

def setup_inputs():
    return {"x": np.random.randn(131072, 1024).astype(np.float32)}

def reference(x: np.ndarray) -> np.ndarray:
    return x
```

```python
import jax
import jax.numpy as jnp
import numpy as np
from jax import lax
from jax.experimental import pallas as pl
from jax.experimental.pallas import tpu as pltpu

SHARD_ROWS = 65536
COLS = 1024

ROWS = 256
STREAM_WORDS = 16
BAND = 8
N_IN = 2
N_OUT = 2
N_SEND = 3
N_RECV_Y = 4
N_RECV_X = 3
VMEM_PIECE_MIB = 112
HBM_PIECES_MIB = (18,) * 8

N_CHUNKS = SHARD_ROWS // 2 // ROWS
N_ITERS = ROWS // 32
RAW_VREGS = ROWS // 2
PACKED_VREGS = STREAM_WORDS + 9 * N_ITERS
PIECE_ROWS = tuple(int(m * 512) for m in (VMEM_PIECE_MIB,) + HBM_PIECES_MIB)
assert sum(PIECE_ROWS) == 2 * SHARD_ROWS

I32 = jnp.int32
BF16 = jnp.bfloat16
MESH = pl.DeviceIdType.MESH
shr = lax.shift_right_logical
shl = lax.shift_left


def c32(v):
    return np.uint32(v & 0xFFFFFFFF).astype(np.int32)


def band_base(group):
    return jnp.clip(shr(group * 214, 10) - (BAND // 2 - 1), 0, STREAM_WORDS - BAND)


def encode(x_ref, loc_ref, msg_ref):
    w0 = pltpu.bitcast(x_ref[0:16, :].astype(BF16), I32)
    mean_magnitude = shr(jnp.sum((w0 & 0x7FFF) + (shr(w0, 16) & 0x7FFF)), 14)
    bias = (mean_magnitude + (4 + 511) + 0x8000) * 0x10001
    zero = jnp.zeros((8, 128), I32)
    top = jnp.full((8, 128), c32(0x80000000), I32)
    for i in range(STREAM_WORDS):
        msg_ref[i] = zero

    def body(t, carry):
        acc, off, word_idx, bad = carry
        r0 = pl.multiple_of(t * 32, 32)
        signs = None
        for s in range(4):
            rows, cols = pl.ds(r0 + 16 * (s // 2), 16), pl.ds(512 * (s % 2), 512)
            b = x_ref[rows, cols].astype(BF16)
            loc_ref[rows, cols] = b
            w = bias - pltpu.bitcast(b, I32)
            for h in range(2):
                ta = w[:, 256 * h : 256 * h + 128]
                tb = w[:, 256 * h + 128 : 256 * h + 256]
                lo = (ta & c32(0x00FF00FF)) | (shl(tb, 8) & c32(0xFF00FF00))
                hi = (shr(ta, 8) & c32(0x00FF00FF)) | (tb & c32(0xFF00FF00))
                msg_ref[STREAM_WORDS + 9 * t + 2 * s + h] = lo
                bad = bad | (hi & c32(0x70707070))
                sg = hi & c32(0x80808080)
                signs = sg if signs is None else (shr(signs, 1) | sg)
                d = hi & c32(0x0F0F0F0F)
                ge4 = (d + c32(0x7C7C7C7C)) & c32(0x80808080)
                lt4 = ge4 ^ c32(0x80808080)
                rank = (d + shr(lt4, 6) + shr(lt4, 7)) & (shr(ge4, 5) | c32(0xFBFBFBFB))
                p = rank + c32(0x01010100)
                p = p + shl(p, 8)
                p = p + shl(p, 16)
                p3 = shr(p, 24)
                bad = bad | shr(p3, 5)
                p3 = p3 & 31
                code = (
                    shr(top, p & 31)
                    | shr(top, shr(p, 8) & 31)
                    | shr(top, shr(p, 16) & 31)
                    | shr(top, p3)
                )
                word = acc | shr(code, off)
                base = band_base(t * 8 + 2 * s + h)
                rel = word_idx - base
                bad = bad | shr(rel, 3)
                for i in range(BAND):
                    pltpu.store(msg_ref.at[base + i], word, mask=rel == i)
                end = off + p3 + 1
                full = shr(end, 5)
                acc = jnp.where(full != 0, shl(shl(code, 1), 31 - off), word)
                off = end & 31
                word_idx = word_idx + full
        msg_ref[STREAM_WORDS + 9 * t + 8] = signs
        return acc, off, word_idx, bad

    acc, off, word_idx, bad = lax.fori_loop(0, N_ITERS, body, (zero,) * 4)
    rel = word_idx - (STREAM_WORDS - BAND)
    for i in range(BAND):
        pltpu.store(msg_ref.at[STREAM_WORDS - BAND + i], acc, mask=rel == i)
    bad = bad | jnp.where((off != 0) & (shr(rel, 3) != 0), 1, 0)
    raw = jnp.max(jnp.where(bad != 0, 1, 0))

    @pl.when(raw != 0)
    def _():
        def copy(t, _):
            w = pltpu.bitcast(loc_ref[pl.ds(pl.multiple_of(t * 16, 16), 16), :], I32)
            for c in range(8):
                msg_ref[t * 8 + c] = w[:, 128 * c : 128 * (c + 1)]

        lax.fori_loop(0, ROWS // 16, copy, None)

    return bias, raw


def decode(msg_ref, out_ref, bias, raw):
    @pl.when(raw != 0)
    def _():
        def copy(t, _):
            w = jnp.concatenate([msg_ref[t * 8 + c] for c in range(8)], axis=1)
            out_ref[pl.ds(pl.multiple_of(t * 16, 16), 16), :] = pltpu.bitcast(w, BF16)

        lax.fori_loop(0, ROWS // 16, copy, None)

    @pl.when(raw == 0)
    def _():
        top = jnp.full((8, 128), c32(0x80000000), I32)

        def body(t, pos):
            r0 = pl.multiple_of(t * 32, 32)
            signs = msg_ref[STREAM_WORDS + 9 * t + 8]
            for s in range(4):
                base = band_base(t * 8 + 2 * s)
                rel = shr(pos, 5) - base
                off = pos & 31
                cand = [msg_ref[base + i] for i in range(BAND + 2)]
                for bit in (4, 2, 1):
                    m = (rel & bit) != 0
                    cand = [jnp.where(m, cand[i + bit], cand[i]) for i in range(bit + 2)]
                a, b, c = cand
                win = shl(a, off) | shr(shr(b, 1), 31 - off)
                nxt = shl(b, off) | shr(shr(c, 1), 31 - off)
                words = []
                for h in range(2):
                    p0 = lax.clz(win)
                    rest = win ^ shr(top, p0)
                    p1 = lax.clz(rest)
                    rest = rest ^ shr(top, p1)
                    p2 = lax.clz(rest)
                    rest = rest ^ shr(top, p2)
                    p3 = lax.clz(rest)
                    if h == 0:
                        win = shl(shl(win, 1), p3) | shr(nxt, 31 - p3)
                    pos = pos + p3 + 1
                    p = p0 | shl(p1, 8) | shl(p2, 16) | shl(p3, 24)
                    rank = p - shl(p, 8) - c32(0x01010100)
                    ge4 = (rank + c32(0x7C7C7C7C)) & c32(0x80808080)
                    lt4 = ge4 ^ c32(0x80808080)
                    d = (rank + shr(lt4, 7)) & (shr(ge4, 5) | c32(0xFBFBFBFB))
                    up = 7 - (2 * s + h)
                    hi = d | ((shl(signs, up) if up else signs) & c32(0x80808080))
                    lo = msg_ref[STREAM_WORDS + 9 * t + 2 * s + h]
                    ta = (lo & c32(0x00FF00FF)) | (shl(hi, 8) & c32(0xFF00FF00))
                    tb = (shr(lo, 8) & c32(0x00FF00FF)) | (hi & c32(0xFF00FF00))
                    words += [bias - ta, bias - tb]
                rows, cols = pl.ds(r0 + 16 * (s // 2), 16), pl.ds(512 * (s % 2), 512)
                out_ref[rows, cols] = pltpu.bitcast(jnp.concatenate(words, axis=1), BF16)
            return pos

        lax.fori_loop(0, N_ITERS, body, jnp.zeros((8, 128), I32))


def all_gather_kernel(x_ref, *refs):
    outs = refs[: len(PIECE_ROWS)]
    (
        in_s, in_o, loc_s, loc_o, dec_y, dec_x,
        snd, rcv_y, rcv_x, hdr_s, hdr_y, hdr_x,
        in_s_sem, in_o_sem, loc_s_sem, loc_o_sem, dec_y_sem, dec_x_sem,
        ys_sem, yr_sem, xs_sem, xr_sem, y_credit, x_credit,
    ) = refs[len(PIECE_ROWS) :]

    my_x, my_y = lax.axis_index("x"), lax.axis_index("y")
    y_peer, x_peer = (my_x, 1 - my_y), (1 - my_x, my_y)
    half = SHARD_ROWS // 2
    send_row = my_x * half
    keep_row = (1 - my_x) * half
    own_row = my_y * SHARD_ROWS
    other_row = (1 - my_y) * SHARD_ROWS

    def load(buf, sem, row, c):
        slot = c % N_IN
        rows = pl.ds(pl.multiple_of(row + c * ROWS, ROWS), ROWS)
        return pltpu.make_async_copy(x_ref.at[rows], buf.at[slot], sem.at[slot])

    def store_start(buf, sem, row, c):
        slot = c % N_OUT
        row = row + c * ROWS
        start = 0
        for out, n in zip(outs, PIECE_ROWS):

            @pl.when((row >= start) & (row < start + n))
            def _(out=out, start=start):
                rows = pl.ds(pl.multiple_of(row - start, ROWS), ROWS)
                pltpu.make_async_copy(buf.at[slot], out.at[rows], sem.at[slot]).start()

            start += n

    def store_wait(buf, sem, c):
        slot = c % N_OUT
        pltpu.make_async_copy(buf.at[slot], buf.at[slot], sem.at[slot]).wait()

    def message(src, src_hdr, send_sem, dst, dst_hdr, recv_sem, peer, c):
        i, j = c % src.shape[0], c % dst.shape[0]
        parts = (
            (src_hdr.at[i], dst_hdr.at[j]),
            (src.at[i, :PACKED_VREGS], dst.at[j, :PACKED_VREGS]),
            (src.at[i, PACKED_VREGS:], dst.at[j, PACKED_VREGS:]),
        )
        return [
            pltpu.make_async_remote_copy(
                s, d, send_sem.at[i, n], recv_sem.at[j, n],
                device_id=peer, device_id_type=MESH,
            )
            for n, (s, d) in enumerate(parts)
        ]

    def y_message(c):
        return message(snd, hdr_s, ys_sem, rcv_y, hdr_y, yr_sem, y_peer, c)

    def x_message(c):
        return message(rcv_y, hdr_y, xs_sem, rcv_x, hdr_x, xr_sem, x_peer, c)

    def send(copies, raw):
        copies[0].start()
        copies[1].start()
        pl.when(raw != 0)(copies[2].start)

    def wait_sent(copies, raw):
        copies[0].wait_send()
        copies[1].wait_send()
        pl.when(raw != 0)(copies[2].wait_send)

    def wait_received(copies, hdr, c):
        copies[0].wait_recv()
        copies[1].wait_recv()
        pl.when(hdr[c % hdr.shape[0], 1] != 0)(copies[2].wait_recv)

    barrier = pltpu.get_barrier_semaphore()
    for peer in (y_peer, x_peer):
        pl.semaphore_signal(barrier, inc=1, device_id=peer, device_id_type=MESH)
    for c in range(N_IN):
        load(in_s, in_s_sem, send_row, c).start()
    for c in range(N_IN):
        load(in_o, in_o_sem, keep_row, c).start()

    def period(c, _):
        @pl.when(c < N_CHUNKS)
        def _():
            slot = c % N_SEND

            @pl.when(c >= N_SEND)
            def _():
                wait_sent(y_message(c - N_SEND), hdr_s[slot, 1])

            pl.when(c >= N_OUT)(lambda: store_wait(loc_s, loc_s_sem, c))
            load(in_s, in_s_sem, send_row, c).wait()
            bias, raw = encode(in_s.at[c % N_IN], loc_s.at[c % N_OUT], snd.at[slot])
            hdr_s[slot, 0] = bias
            hdr_s[slot, 1] = raw
            pl.when(c == 0)(lambda: pl.semaphore_wait(barrier, 2))
            pl.when(c >= N_RECV_Y)(
                lambda: pl.semaphore_wait(y_credit.at[c % N_RECV_Y], 1)
            )
            send(y_message(c), raw)
            store_start(loc_s, loc_s_sem, own_row + send_row, c)
            pl.when(c + N_IN < N_CHUNKS)(
                lambda: load(in_s, in_s_sem, send_row, c + N_IN).start()
            )

            pl.when(c >= N_OUT)(lambda: store_wait(loc_o, loc_o_sem, c))
            load(in_o, in_o_sem, keep_row, c).wait()

            def convert(t, _):
                rows = pl.ds(pl.multiple_of(t * 32, 32), 32)
                loc_o[c % N_OUT, rows, :] = in_o[c % N_IN, rows, :].astype(BF16)

            lax.fori_loop(0, ROWS // 32, convert, None)
            store_start(loc_o, loc_o_sem, own_row + keep_row, c)
            pl.when(c + N_IN < N_CHUNKS)(
                lambda: load(in_o, in_o_sem, keep_row, c + N_IN).start()
            )

        @pl.when(c >= 3)
        def _():
            cx = c - 3
            slot = cx % N_RECV_X
            wait_received(x_message(cx), hdr_x, cx)
            pl.when(cx >= N_OUT)(lambda: store_wait(dec_x, dec_x_sem, cx))
            decode(rcv_x.at[slot], dec_x.at[cx % N_OUT], hdr_x[slot, 0], hdr_x[slot, 1])
            store_start(dec_x, dec_x_sem, other_row + keep_row, cx)

            @pl.when(cx + N_RECV_X < N_CHUNKS)
            def _():
                pl.semaphore_signal(
                    x_credit.at[slot], inc=1, device_id=x_peer, device_id_type=MESH
                )

            wait_sent(x_message(cx), hdr_y[cx % N_RECV_Y, 1])

            @pl.when(cx + N_RECV_Y < N_CHUNKS)
            def _():
                pl.semaphore_signal(
                    y_credit.at[cx % N_RECV_Y],
                    inc=1,
                    device_id=y_peer,
                    device_id_type=MESH,
                )

        @pl.when((c >= 2) & (c < N_CHUNKS + 2))
        def _():
            cy = c - 2
            slot = cy % N_RECV_Y
            pl.when(cy >= N_OUT)(lambda: store_wait(dec_y, dec_y_sem, cy))
            decode(rcv_y.at[slot], dec_y.at[cy % N_OUT], hdr_y[slot, 0], hdr_y[slot, 1])
            store_start(dec_y, dec_y_sem, other_row + send_row, cy)

        @pl.when((c >= 1) & (c < N_CHUNKS + 1))
        def _():
            k = c - 1
            pl.when(k >= N_RECV_X)(
                lambda: pl.semaphore_wait(x_credit.at[k % N_RECV_X], 1)
            )
            wait_received(y_message(k), hdr_y, k)
            send(x_message(k), hdr_y[k % N_RECV_Y, 1])

    lax.fori_loop(0, N_CHUNKS + 3, period, None)

    for c in range(N_CHUNKS - N_SEND, N_CHUNKS):
        wait_sent(y_message(c), hdr_s[c % N_SEND, 1])
    for c in range(N_CHUNKS - N_OUT, N_CHUNKS):
        store_wait(loc_s, loc_s_sem, c)
        store_wait(loc_o, loc_o_sem, c)
        store_wait(dec_y, dec_y_sem, c)
        store_wait(dec_x, dec_x_sem, c)


def pallas_dist_ag_xy_y_m65536_n1024_kernel(x: jax.Array):
    assert x.shape == (SHARD_ROWS, COLS) and x.dtype == jnp.float32
    dma = pltpu.SemaphoreType.DMA
    pieces = pl.pallas_call(
        all_gather_kernel,
        out_shape=(pltpu.VMEM((PIECE_ROWS[0], COLS), BF16),)
        + tuple(jax.ShapeDtypeStruct((n, COLS), BF16) for n in PIECE_ROWS[1:]),
        in_specs=[pl.BlockSpec(memory_space=pl.ANY)],
        out_specs=(pl.BlockSpec(memory_space=pltpu.VMEM),)
        + (pl.BlockSpec(memory_space=pl.ANY),) * (len(PIECE_ROWS) - 1),
        scratch_shapes=[
            pltpu.VMEM((N_IN, ROWS, COLS), jnp.float32),
            pltpu.VMEM((N_IN, ROWS, COLS), jnp.float32),
            pltpu.VMEM((N_OUT, ROWS, COLS), BF16),
            pltpu.VMEM((N_OUT, ROWS, COLS), BF16),
            pltpu.VMEM((N_OUT, ROWS, COLS), BF16),
            pltpu.VMEM((N_OUT, ROWS, COLS), BF16),
            pltpu.VMEM((N_SEND, RAW_VREGS, 8, 128), I32),
            pltpu.VMEM((N_RECV_Y, RAW_VREGS, 8, 128), I32),
            pltpu.VMEM((N_RECV_X, RAW_VREGS, 8, 128), I32),
            pltpu.SMEM((N_SEND, 2), I32),
            pltpu.SMEM((N_RECV_Y, 2), I32),
            pltpu.SMEM((N_RECV_X, 2), I32),
            dma((N_IN,)),
            dma((N_IN,)),
            dma((N_OUT,)),
            dma((N_OUT,)),
            dma((N_OUT,)),
            dma((N_OUT,)),
            dma((N_SEND, 3)),
            dma((N_RECV_Y, 3)),
            dma((N_RECV_Y, 3)),
            dma((N_RECV_X, 3)),
            pltpu.SemaphoreType.REGULAR((N_RECV_Y,)),
            pltpu.SemaphoreType.REGULAR((N_RECV_X,)),
        ],
        compiler_params=pltpu.CompilerParams(collective_id=0),
    )(x)
    return jnp.concatenate(pieces, axis=0)
```

```python
import functools

import jax
import jax.numpy as jnp
import numpy as np
from jax import lax
from jax.experimental import pallas as pl
from jax.experimental.pallas import tpu as pltpu

SHARD_ROWS = 65536
COLS = 1024

TICK_ROWS = 128
TICKS = 4
STREAM_WORDS = 30
DENSE_WORDS = 26
BAND = 8
TOP_OFFSET = 452

FORWARD_LAG = 2
DECODE_LAG = 6
N_IN = 2
N_OUT = 2
N_SEND = 2
N_RECV = 3
VMEM_PIECES_MIB = (84, 14, 14)
HBM_PIECES_MIB = (60, 84)

CHUNK_ROWS = TICKS * TICK_ROWS
N_TICKS = SHARD_ROWS // 2 // TICK_ROWS
N_CHUNKS = N_TICKS // TICKS
TICK_ITERS = TICK_ROWS // 32
PLANE_VREGS = 9 * TICK_ITERS
STREAM_AT = TICKS * PLANE_VREGS
BINADES_AT = STREAM_AT + STREAM_WORDS
SLOT_VREGS = BINADES_AT + TICKS * 8 * TICK_ITERS
PIECE_ROWS = tuple(int(m * 512) for m in VMEM_PIECES_MIB + HBM_PIECES_MIB)
assert sum(PIECE_ROWS) == 2 * SHARD_ROWS

I32 = jnp.int32
BF16 = jnp.bfloat16
MESH = pl.DeviceIdType.MESH
HEADER, STREAMS, BINADES, PLANES = range(4)
shr = lax.shift_right_logical
shl = lax.shift_left


def c32(v):
    return np.uint32(v & 0xFFFFFFFF).astype(np.int32)


def at_least(x, k):
    return shr(x + c32(0x01010101 * (128 - k)), 7) & c32(0x01010101)


def band_base(group):
    typical = shr(group * 209 + 768, 10)
    return jnp.clip(typical - BAND // 2, 0, STREAM_WORDS - BAND)


def lane_counts(flags, counter_ref):
    ones = jnp.where(flags, 1.0, 0.0).astype(BF16)
    counts = jnp.dot(ones, counter_ref[...], preferred_element_type=jnp.float32)
    counts = counts.astype(I32)
    return counts[:, :128], counts[:, 128:]


def store_word(msg_ref, base, word_idx, word):
    rel = word_idx - base
    for i in range(BAND):
        pltpu.store(msg_ref.at[STREAM_AT + base + i], word, mask=rel == i)
    return shr(rel, 3)


def encode_begin(x_ref, msg_ref, state_ref):
    w = pltpu.bitcast(x_ref[0:16, :].astype(BF16), I32)
    mean_magnitude = shr(jnp.sum((w & 0x7FFF) + (shr(w, 16) & 0x7FFF)), 14)
    zero = jnp.zeros((8, 128), I32)
    for i in range(STREAM_WORDS):
        msg_ref[STREAM_AT + i] = zero
    for i in range(state_ref.shape[0]):
        state_ref[i] = zero
    return (mean_magnitude + TOP_OFFSET + 0x8000) * 0x10001


def encode_rows(x_ref, loc_ref, msg_ref, state_ref, bias, tick):
    top = jnp.full((8, 128), c32(0x80000000), I32)

    def body(i, carry):
        acc, off, word_idx, bad, binades = carry
        t = tick * TICK_ITERS + i
        odd = None
        for s in range(4):
            rows = pl.ds(pl.multiple_of(i * 32, 32) + 16 * (s // 2), 16)
            cols = pl.ds(512 * (s % 2), 512)
            b = x_ref[rows, cols].astype(BF16)
            loc_ref[rows, cols] = b
            w = bias - pltpu.bitcast(b, I32)
            for h in range(2):
                g = 2 * s + h
                ta = w[:, 256 * h : 256 * h + 128]
                tb = w[:, 256 * h + 128 : 256 * h + 256]
                msg_ref[9 * t + g] = (
                    (ta & c32(0x007F007F))
                    | (shr(ta, 8) & c32(0x00800080))
                    | (shl(tb, 8) & c32(0x7F007F00))
                    | (tb & c32(0x80008000))
                )
                d = (shr(ta, 7) & c32(0x00FF00FF)) | (shl(tb, 1) & c32(0xFF00FF00))
                msg_ref[BINADES_AT + 8 * t + g] = d
                binades = binades | d
                ge4 = at_least(d, 4)
                n = (d ^ ((ge4 ^ c32(0x01010101)) * 3)) - ge4 + at_least(d, 10)
                n = n + c32(0x06060606) - at_least(d, 1) * 6
                last = n & c32(0x01010101)
                odd = last if odd is None else (shl(odd, 1) | last)
                p = (shr(n, 1) & c32(0x0F0F0F0F)) + c32(0x01010100)
                p = p * c32(0x01010101)
                p3 = shr(p, 24)
                bad = bad | shr(p3, 5)
                p3 = p3 & 31
                code = (
                    shr(top, p & 31)
                    | shr(top, shr(p, 8) & 31)
                    | shr(top, shr(p, 16) & 31)
                    | shr(top, p3)
                )
                word = acc | shr(code, off)
                bad = bad | store_word(msg_ref, band_base(8 * t + g), word_idx, word)
                end = off + p3 + 1
                full = shr(end, 5)
                acc = jnp.where(full != 0, shl(shl(code, 1), 31 - off), word)
                off = end & 31
                word_idx = word_idx + full
        msg_ref[9 * t + 8] = odd
        return acc, off, word_idx, bad, binades

    state = tuple(state_ref[i] for i in range(state_ref.shape[0]))
    state = lax.fori_loop(0, TICK_ITERS, body, state)
    for i, value in enumerate(state):
        state_ref[i] = value


def encode_end(msg_ref, state_ref, counter_ref):
    acc, off, word_idx, bad, binades = (state_ref[i] for i in range(5))
    lost = store_word(msg_ref, STREAM_WORDS - BAND, word_idx, acc)
    bad = bad | jnp.where(off != 0, lost, 0) | (binades & c32(0xE0E0E0E0))

    n_words = word_idx + jnp.where(off != 0, 1, 0)
    pooled = range(DENSE_WORDS, STREAM_WORDS)
    used = jnp.concatenate([n_words > i for i in pooled], axis=0)
    before, total = lane_counts(used, counter_ref)
    lane = lax.broadcasted_iota(I32, used.shape, 1)
    val = jnp.concatenate([msg_ref[STREAM_AT + i] for i in pooled], axis=0)
    move = jnp.where(used, lane - before, 0)
    for k in (1, 2, 4, 8, 16, 32, 64):
        val_in, move_in = pltpu.roll(val, 128 - k, 1), pltpu.roll(move, 128 - k, 1)
        take = (move_in & k) != 0
        val = jnp.where(take, val_in, val)
        move = jnp.where(take, move_in, jnp.where((move & k) != 0, 0, move))
    pool, filled = val[0:8], total[0:8]
    for i in range(1, len(pooled)):
        slot = lane[0:8] - filled
        more = jnp.take_along_axis(val[8 * i : 8 * i + 8], slot & 127, axis=1)
        pool = jnp.where(slot < 0, pool, more)
        filled = filled + total[8 * i : 8 * i + 8]
    msg_ref[STREAM_AT + DENSE_WORDS] = pool
    bad = bad | jnp.where(filled > 128, 1, 0)
    return jnp.max(jnp.where(bad != 0, 1, 0))


def decode_begin(msg_ref, stream_ref, pos_ref, counter_ref):
    markers = []
    for i in range(DENSE_WORDS):
        word = msg_ref[STREAM_AT + i]
        stream_ref[i] = word
        markers.append(lax.population_count(word))
    markers = functools.reduce(jnp.add, markers)
    pool, filled = msg_ref[STREAM_AT + DENSE_WORDS], 0
    for i in range(DENSE_WORDS, STREAM_WORDS):
        used = markers < CHUNK_ROWS
        before, total = lane_counts(used, counter_ref)
        word = jnp.take_along_axis(pool, (filled + before) & 127, axis=1)
        word = jnp.where(used, word, 0)
        stream_ref[i] = word
        markers = markers + lax.population_count(word)
        filled = filled + total
    pos_ref[...] = jnp.zeros((8, 128), I32)


def decode_rows(jobs, tick):
    top = jnp.full((8, 128), c32(0x80000000), I32)

    def step(i, s, job, pos):
        msg_ref, stream_ref, _, out_ref, bias, raw = job
        t = tick * TICK_ITERS + i
        base = band_base(8 * t + 2 * s)
        rel = shr(pos, 5) - base
        off = pos & 31
        cand = [
            stream_ref[base + k if k < BAND else jnp.minimum(base + k, STREAM_WORDS - 1)]
            for k in range(BAND + 2)
        ]
        for bit in (4, 2, 1):
            m = (rel & bit) != 0
            cand = [jnp.where(m, cand[k + bit], cand[k]) for k in range(bit + 2)]
        a, b, c = cand
        win = shl(a, off) | shr(shr(b, 1), 31 - off)
        nxt = shl(b, off) | shr(shr(c, 1), 31 - off)
        odd = msg_ref[9 * t + 8]
        words = []
        for h in range(2):
            g = 2 * s + h
            p0 = lax.clz(win)
            rest = win ^ shr(top, p0)
            p1 = lax.clz(rest)
            rest = rest ^ shr(top, p1)
            p2 = lax.clz(rest)
            rest = rest ^ shr(top, p2)
            p3 = lax.clz(rest)
            if h == 0:
                win = shl(shl(win, 1), p3) | shr(nxt, 31 - p3)
            pos = pos + p3 + 1
            p = p0 | shl(p1, 8) | shl(p2, 16) | shl(p3, 24)
            n = p * c32(2 - 512) - c32(0x02020200)
            n = n | ((shr(odd, 7 - g) if g < 7 else odd) & c32(0x01010101))
            ge3 = at_least(n, 3)
            d = (n ^ ((ge3 ^ c32(0x01010101)) * 3)) + ge3
            d = d + at_least(n, 10) * 9 - at_least(n, 9) * 10
            d = jnp.where(raw != 0, msg_ref[BINADES_AT + 8 * t + g], d)
            low = msg_ref[9 * t + g]
            ta = (
                (low & c32(0x007F007F))
                | (shl(low, 8) & c32(0x80008000))
                | (shl(d, 7) & c32(0x7F807F80))
            )
            tb = (
                (shr(low, 8) & c32(0x007F007F))
                | (low & c32(0x80008000))
                | (shr(d, 1) & c32(0x7F807F80))
            )
            words += [bias - ta, bias - tb]
        rows = pl.ds(pl.multiple_of(i * 32, 32) + 16 * (s // 2), 16)
        cols = pl.ds(512 * (s % 2), 512)
        out_ref[rows, cols] = pltpu.bitcast(jnp.concatenate(words, axis=1), BF16)
        return pos

    def body(i, positions):
        for s in range(4):
            positions = tuple(step(i, s, j, p) for j, p in zip(jobs, positions))
        return positions

    positions = tuple(job[2][...] for job in jobs)
    positions = lax.fori_loop(0, TICK_ITERS, body, positions)
    for job, pos in zip(jobs, positions):
        job[2][...] = pos


def all_gather_kernel(x_ref, *refs):
    outs = refs[: len(PIECE_ROWS)]
    (
        in_s, in_k, loc_s, loc_k, dec_y, dec_x,
        msg_s, msg_y, msg_x, hdr_s, hdr_y, hdr_x,
        enc_state, dec_stream, dec_pos, counter,
        in_s_sem, in_k_sem, loc_s_sem, loc_k_sem, dec_y_sem, dec_x_sem,
        y_sent, y_landed, x_sent, x_landed, y_credit, x_credit,
    ) = refs[len(PIECE_ROWS) :]

    my_x, my_y = lax.axis_index("x"), lax.axis_index("y")
    y_peer, x_peer = (my_x, 1 - my_y), (1 - my_x, my_y)
    send_row = my_x * (SHARD_ROWS // 2)
    keep_row = (1 - my_x) * (SHARD_ROWS // 2)
    own_row = my_y * SHARD_ROWS
    other_row = (1 - my_y) * SHARD_ROWS

    def load(buf, sem, row, tick):
        slot = tick % N_IN
        rows = pl.ds(pl.multiple_of(row + tick * TICK_ROWS, TICK_ROWS), TICK_ROWS)
        return pltpu.make_async_copy(x_ref.at[rows], buf.at[slot], sem.at[slot])

    def load_ahead(buf, sem, row, tick):
        @pl.when(tick + N_IN < N_TICKS)
        def _():
            load(buf, sem, row, tick + N_IN).start()

    def store(buf, sem, row, tick):
        slot = tick % N_OUT
        row = row + tick * TICK_ROWS
        start = 0
        for out, n in zip(outs, PIECE_ROWS):

            @pl.when((row >= start) & (row < start + n))
            def _(out=out, start=start):
                rows = pl.ds(pl.multiple_of(row - start, TICK_ROWS), TICK_ROWS)
                pltpu.make_async_copy(buf.at[slot], out.at[rows], sem.at[slot]).start()

            start += n

    def wait_stored(buf, sem, tick):
        slot = tick % N_OUT
        pltpu.make_async_copy(buf.at[slot], buf.at[slot], sem.at[slot]).wait()

    def copy(src, dst, peer, chunk, kind, half):
        (src_hdr, src_msg, sent), (dst_hdr, dst_msg, landed) = src, dst
        i, j = chunk % src_msg.shape[0], chunk % dst_msg.shape[0]
        if kind == HEADER:
            a, b = src_hdr.at[i], dst_hdr.at[j]
        else:
            part = {
                STREAMS: pl.ds(STREAM_AT, DENSE_WORDS + 1),
                BINADES: pl.ds(BINADES_AT, SLOT_VREGS - BINADES_AT),
                PLANES: pl.ds(half * (PLANE_VREGS // 2), PLANE_VREGS // 2),
            }[kind]
            a, b = src_msg.at[i, part], dst_msg.at[j, part]
        return pltpu.make_async_remote_copy(
            a, b, sent.at[i, kind + half], landed.at[j, kind + half],
            device_id=peer, device_id_type=MESH,
        )

    def over_y(chunk, kind, half=0):
        src, dst = (hdr_s, msg_s, y_sent), (hdr_y, msg_y, y_landed)
        return copy(src, dst, y_peer, chunk, kind, half)

    def over_x(chunk, kind, half=0):
        src, dst = (hdr_y, msg_y, x_sent), (hdr_x, msg_x, x_landed)
        return copy(src, dst, x_peer, chunk, kind, half)

    def wait_tail_sent(link, chunk, raw):
        link(chunk, HEADER).wait_send()
        link(chunk, STREAMS).wait_send()
        pl.when(raw != 0)(lambda: link(chunk, BINADES).wait_send())

    def send_own(tick):
        chunk, j = tick // TICKS, tick % TICKS
        slot = chunk % N_SEND

        @pl.when(chunk >= N_SEND)
        def _():
            old = chunk - N_SEND
            pl.when(j == 0)(lambda: wait_tail_sent(over_y, old, hdr_s[slot, 1]))
            over_y(old, PLANES, 2 * j).wait_send()
            over_y(old, PLANES, 2 * j + 1).wait_send()

        pl.when(tick >= N_OUT)(lambda: wait_stored(loc_s, loc_s_sem, tick))
        load(in_s, in_s_sem, send_row, tick).wait()

        @pl.when(tick == 0)
        def _():
            for i in range(1, N_IN):
                load(in_s, in_s_sem, send_row, i).start()
            for i in range(N_IN):
                load(in_k, in_k_sem, keep_row, i).start()

        x, msg = in_s.at[tick % N_IN], msg_s.at[slot]

        @pl.when(j == 0)
        def _():
            hdr_s[slot, 0] = encode_begin(x, msg, enc_state)

        encode_rows(x, loc_s.at[tick % N_OUT], msg, enc_state, hdr_s[slot, 0], j)
        pl.when(tick == 0)(lambda: pl.semaphore_wait(barrier, 2))
        pl.when((j == 0) & (chunk >= N_RECV))(
            lambda: pl.semaphore_wait(y_credit.at[chunk % N_RECV], 1)
        )

        @pl.when(j == TICKS - 1)
        def _():
            raw = encode_end(msg, enc_state, counter)
            hdr_s[slot, 1] = raw
            over_y(chunk, HEADER).start()
            over_y(chunk, STREAMS).start()
            pl.when(raw != 0)(lambda: over_y(chunk, BINADES).start())

        over_y(chunk, PLANES, 2 * j).start()
        over_y(chunk, PLANES, 2 * j + 1).start()
        store(loc_s, loc_s_sem, own_row + send_row, tick)
        load_ahead(in_s, in_s_sem, send_row, tick)

    def keep_own(tick):
        pl.when(tick >= N_OUT)(lambda: wait_stored(loc_k, loc_k_sem, tick))
        load(in_k, in_k_sem, keep_row, tick).wait()
        loc_k[tick % N_OUT] = in_k[tick % N_IN].astype(BF16)
        store(loc_k, loc_k_sem, own_row + keep_row, tick)
        load_ahead(in_k, in_k_sem, keep_row, tick)

    def forward(tick, h):
        chunk, j = tick // TICKS, tick % TICKS

        def relay(kind, half=0):
            over_y(chunk, kind, half).wait_recv()
            over_x(chunk, kind, half).start()

        if h == 0:
            pl.when((j == 0) & (chunk >= N_RECV))(
                lambda: pl.semaphore_wait(x_credit.at[chunk % N_RECV], 1)
            )

            @pl.when(j == TICKS - 1)
            def _():
                relay(HEADER)
                relay(STREAMS)
                pl.when(hdr_y[chunk % N_RECV, 1] != 0)(lambda: relay(BINADES))

        relay(PLANES, 2 * j + h)

    def receive(tick):
        chunk, j = tick // TICKS, tick % TICKS
        slot, o = chunk % N_RECV, tick % N_OUT

        @pl.when(j == 0)
        def _():
            over_x(chunk, HEADER).wait_recv()
            over_x(chunk, STREAMS).wait_recv()
            pl.when(hdr_x[slot, 1] != 0)(lambda: over_x(chunk, BINADES).wait_recv())
            decode_begin(msg_y.at[slot], dec_stream.at[0], dec_pos.at[0], counter)
            decode_begin(msg_x.at[slot], dec_stream.at[1], dec_pos.at[1], counter)

        over_x(chunk, PLANES, 2 * j).wait_recv()
        over_x(chunk, PLANES, 2 * j + 1).wait_recv()
        pl.when(tick >= N_OUT)(lambda: wait_stored(dec_y, dec_y_sem, tick))
        pl.when(tick >= N_OUT)(lambda: wait_stored(dec_x, dec_x_sem, tick))
        decode_rows(
            [
                (msg.at[slot], dec_stream.at[k], dec_pos.at[k], out.at[o], hdr[slot, 0], hdr[slot, 1])
                for k, (msg, hdr, out) in enumerate(((msg_y, hdr_y, dec_y), (msg_x, hdr_x, dec_x)))
            ],
            j,
        )
        store(dec_y, dec_y_sem, other_row + send_row, tick)
        store(dec_x, dec_x_sem, other_row + keep_row, tick)
        over_x(chunk, PLANES, 2 * j).wait_send()
        over_x(chunk, PLANES, 2 * j + 1).wait_send()

        @pl.when(j == TICKS - 1)
        def _():
            wait_tail_sent(over_x, chunk, hdr_y[slot, 1])

            @pl.when(chunk + N_RECV < N_CHUNKS)
            def _():
                for credit, peer in ((y_credit, y_peer), (x_credit, x_peer)):
                    pl.semaphore_signal(credit.at[slot], inc=1, device_id=peer, device_id_type=MESH)

    barrier = pltpu.get_barrier_semaphore()
    load(in_s, in_s_sem, send_row, 0).start()
    for peer in (y_peer, x_peer):
        pl.semaphore_signal(barrier, inc=1, device_id=peer, device_id_type=MESH)
    r = lax.broadcasted_iota(I32, (128, 256), 0)
    q = lax.broadcasted_iota(I32, (128, 256), 1)
    counter[...] = jnp.where(r < q, 1.0, 0.0).astype(BF16)

    def run_tick(tick, _):
        relayed = tick - FORWARD_LAG
        relaying = (tick >= FORWARD_LAG) & (tick < N_TICKS + FORWARD_LAG)
        pl.when(tick < N_TICKS)(lambda: send_own(tick))
        pl.when(relaying)(lambda: forward(relayed, 0))
        pl.when(tick < N_TICKS)(lambda: keep_own(tick))
        pl.when(tick >= DECODE_LAG)(lambda: receive(tick - DECODE_LAG))
        pl.when(relaying)(lambda: forward(relayed, 1))

    lax.fori_loop(0, N_TICKS + DECODE_LAG, run_tick, None)

    for chunk in range(N_CHUNKS - N_SEND, N_CHUNKS):
        wait_tail_sent(over_y, chunk, hdr_s[chunk % N_SEND, 1])
        for half in range(2 * TICKS):
            over_y(chunk, PLANES, half).wait_send()
    for tick in range(N_TICKS - N_OUT, N_TICKS):
        wait_stored(loc_s, loc_s_sem, tick)
        wait_stored(loc_k, loc_k_sem, tick)
        wait_stored(dec_y, dec_y_sem, tick)
        wait_stored(dec_x, dec_x_sem, tick)


def pallas_dist_ag_xy_y_m65536_n1024_kernel(x: jax.Array):
    assert x.shape == (SHARD_ROWS, COLS) and x.dtype == jnp.float32
    dma = pltpu.SemaphoreType.DMA
    n_vmem = len(VMEM_PIECES_MIB)
    n_copies = PLANES + 2 * TICKS
    pieces = pl.pallas_call(
        all_gather_kernel,
        out_shape=tuple(pltpu.VMEM((n, COLS), BF16) for n in PIECE_ROWS[:n_vmem])
        + tuple(jax.ShapeDtypeStruct((n, COLS), BF16) for n in PIECE_ROWS[n_vmem:]),
        in_specs=[pl.BlockSpec(memory_space=pl.ANY)],
        out_specs=(pl.BlockSpec(memory_space=pltpu.VMEM),) * n_vmem
        + (pl.BlockSpec(memory_space=pl.ANY),) * len(HBM_PIECES_MIB),
        scratch_shapes=[
            *[pltpu.VMEM((N_IN, TICK_ROWS, COLS), jnp.float32)] * 2,
            *[pltpu.VMEM((N_OUT, TICK_ROWS, COLS), BF16)] * 4,
            *[pltpu.VMEM((n, SLOT_VREGS, 8, 128), I32) for n in (N_SEND, N_RECV, N_RECV)],
            *[pltpu.SMEM((n, 2), I32) for n in (N_SEND, N_RECV, N_RECV)],
            pltpu.VMEM((5, 8, 128), I32),
            pltpu.VMEM((2, STREAM_WORDS, 8, 128), I32),
            pltpu.VMEM((2, 8, 128), I32),
            pltpu.VMEM((128, 256), BF16),
            *[dma((N_IN,))] * 2,
            *[dma((N_OUT,))] * 4,
            *[dma((n, n_copies)) for n in (N_SEND, N_RECV, N_RECV, N_RECV)],
            *[pltpu.SemaphoreType.REGULAR((N_RECV,))] * 2,
        ],
        compiler_params=pltpu.CompilerParams(collective_id=0),
    )(x)
    return jnp.concatenate(pieces, axis=0)
```

```python
import functools

import jax
import jax.numpy as jnp
import numpy as np
from jax import lax
from jax.experimental import pallas as pl
from jax.experimental.pallas import tpu as pltpu

SHARD_ROWS = 65536
COLS = 1024

TICK_ROWS = 128
TICKS = 4
STREAM_WORDS = 30
DENSE_WORDS = 26
BAND = 8
TOP_OFFSET = 456

FORWARD_LAG = 2
DECODE_LAG = 6
N_IN = 2
N_OUT = 2
N_SEND = 2
N_RECV = 3
VMEM_TICKS = (447, 1)
STAGED_TICKS = (447, 128)

CHUNK_ROWS = TICKS * TICK_ROWS
N_TICKS = SHARD_ROWS // 2 // TICK_ROWS
N_CHUNKS = N_TICKS // TICKS
TICK_ITERS = TICK_ROWS // 32
PLANE_VREGS = 9 * TICK_ITERS
STREAM_AT = TICKS * PLANE_VREGS
BINADES_AT = STREAM_AT + STREAM_WORDS
SLOT_VREGS = BINADES_AT + TICKS * 8 * TICK_ITERS
PIECE_ROWS = tuple(n * TICK_ROWS for n in VMEM_TICKS)
PIECE_ROWS += (2 * SHARD_ROWS - sum(PIECE_ROWS),)

I32 = jnp.int32
BF16 = jnp.bfloat16
MESH = pl.DeviceIdType.MESH
HEADER, STREAMS, BINADES, PLANES = range(4)
shr = lax.shift_right_logical
shl = lax.shift_left


def c32(v):
    return np.uint32(v & 0xFFFFFFFF).astype(np.int32)


def at_least(x, k):
    return shr(x + c32(0x01010101 * (128 - k)), 7) & c32(0x01010101)


def band_base(group):
    typical = shr(group * 209 + 768, 10)
    return jnp.clip(typical - BAND // 2, 0, STREAM_WORDS - BAND)


def lane_counts(flags, counter_ref):
    ones = jnp.where(flags, 1.0, 0.0).astype(BF16)
    counts = jnp.dot(ones, counter_ref[...], preferred_element_type=jnp.float32)
    counts = counts.astype(I32)
    return counts[:, :128], counts[:, 128:]


def store_word(msg_ref, base, word_idx, word):
    rel = word_idx - base
    for i in range(BAND):
        pltpu.store(msg_ref.at[STREAM_AT + base + i], word, mask=rel == i)
    return shr(rel, 3)


def encode_begin(x_ref, msg_ref, state_ref):
    w = pltpu.bitcast(x_ref[0:16, :].astype(BF16), I32)
    mean_magnitude = shr(jnp.sum((w & 0x7FFF) + (shr(w, 16) & 0x7FFF)), 14)
    zero = jnp.zeros((8, 128), I32)
    for i in range(STREAM_WORDS):
        msg_ref[STREAM_AT + i] = zero
    for i in range(state_ref.shape[0]):
        state_ref[i] = zero
    return (mean_magnitude + TOP_OFFSET + 0x8000) * 0x10001


def encode_rows(x_ref, loc_ref, msg_ref, state_ref, bias, tick):
    top = jnp.full((8, 128), c32(0x80000000), I32)

    def body(i, carry):
        acc, off, word_idx, bad, binades = carry
        t = tick * TICK_ITERS + i
        odd = None
        for s in range(4):
            rows = pl.ds(pl.multiple_of(i * 32, 32) + 16 * (s // 2), 16)
            cols = pl.ds(512 * (s % 2), 512)
            b = x_ref[rows, cols].astype(BF16)
            loc_ref[rows, cols] = b
            w = bias - pltpu.bitcast(b, I32)
            for h in range(2):
                g = 2 * s + h
                ta = w[:, 256 * h : 256 * h + 128]
                tb = w[:, 256 * h + 128 : 256 * h + 256]
                msg_ref[9 * t + g] = (
                    (ta & c32(0x007F007F))
                    | (shr(ta, 8) & c32(0x00800080))
                    | (shl(tb, 8) & c32(0x7F007F00))
                    | (tb & c32(0x80008000))
                )
                d = (shr(ta, 7) & c32(0x00FF00FF)) | (shl(tb, 1) & c32(0xFF00FF00))
                msg_ref[BINADES_AT + 8 * t + g] = d
                binades = binades | d
                ge4 = at_least(d, 4)
                n = (d ^ ((ge4 ^ c32(0x01010101)) * 3)) - ge4 + at_least(d, 10)
                n = n + c32(0x06060606) - at_least(d, 1) * 6
                last = n & c32(0x01010101)
                odd = last if odd is None else (shl(odd, 1) | last)
                p = (shr(n, 1) & c32(0x1F1F1F1F)) + c32(0x01010100)
                p = p * c32(0x01010101)
                p3 = shr(p, 24)
                bad = bad | shr(p3, 5)
                p3 = p3 & 31
                code = (
                    shr(top, p & 31)
                    | shr(top, shr(p, 8) & 31)
                    | shr(top, shr(p, 16) & 31)
                    | shr(top, p3)
                )
                word = acc | shr(code, off)
                bad = bad | store_word(msg_ref, band_base(8 * t + g), word_idx, word)
                end = off + p3 + 1
                full = shr(end, 5)
                acc = jnp.where(full != 0, shl(shl(code, 1), 31 - off), word)
                off = end & 31
                word_idx = word_idx + full
        msg_ref[9 * t + 8] = odd
        return acc, off, word_idx, bad, binades

    state = tuple(state_ref[i] for i in range(state_ref.shape[0]))
    state = lax.fori_loop(0, TICK_ITERS, body, state)
    for i, value in enumerate(state):
        state_ref[i] = value


def encode_end(msg_ref, state_ref, counter_ref):
    acc, off, word_idx, bad, binades = (state_ref[i] for i in range(5))
    lost = store_word(msg_ref, STREAM_WORDS - BAND, word_idx, acc)
    bad = bad | jnp.where(off != 0, lost, 0) | (binades & c32(0xC0C0C0C0))

    n_words = word_idx + jnp.where(off != 0, 1, 0)
    pooled = range(DENSE_WORDS, STREAM_WORDS)
    used = jnp.concatenate([n_words > i for i in pooled], axis=0)
    before, total = lane_counts(used, counter_ref)
    lane = lax.broadcasted_iota(I32, used.shape, 1)
    val = jnp.concatenate([msg_ref[STREAM_AT + i] for i in pooled], axis=0)
    move = jnp.where(used, lane - before, 0)
    for k in (1, 2, 4, 8, 16, 32, 64):
        val_in, move_in = pltpu.roll(val, 128 - k, 1), pltpu.roll(move, 128 - k, 1)
        take = (move_in & k) != 0
        val = jnp.where(take, val_in, val)
        move = jnp.where(take, move_in, jnp.where((move & k) != 0, 0, move))
    pool, filled = val[0:8], total[0:8]
    for i in range(1, len(pooled)):
        slot = lane[0:8] - filled
        more = jnp.take_along_axis(val[8 * i : 8 * i + 8], slot & 127, axis=1)
        pool = jnp.where(slot < 0, pool, more)
        filled = filled + total[8 * i : 8 * i + 8]
    msg_ref[STREAM_AT + DENSE_WORDS] = pool
    bad = bad | jnp.where(filled > 128, 1, 0)
    return jnp.max(jnp.where(bad != 0, 1, 0))


def decode_begin(msg_ref, stream_ref, pos_ref, counter_ref):
    markers = []
    for i in range(DENSE_WORDS):
        word = msg_ref[STREAM_AT + i]
        stream_ref[i] = word
        markers.append(lax.population_count(word))
    markers = functools.reduce(jnp.add, markers)
    pool, filled = msg_ref[STREAM_AT + DENSE_WORDS], 0
    for i in range(DENSE_WORDS, STREAM_WORDS):
        used = markers < CHUNK_ROWS
        before, total = lane_counts(used, counter_ref)
        word = jnp.take_along_axis(pool, (filled + before) & 127, axis=1)
        word = jnp.where(used, word, 0)
        stream_ref[i] = word
        markers = markers + lax.population_count(word)
        filled = filled + total
    pos_ref[...] = jnp.zeros((8, 128), I32)


def decode_rows(jobs, tick):
    top = jnp.full((8, 128), c32(0x80000000), I32)

    def step(i, s, job, pos):
        msg_ref, stream_ref, _, out_ref, bias, raw = job
        t = tick * TICK_ITERS + i
        base = band_base(8 * t + 2 * s)
        rel = shr(pos, 5) - base
        off = pos & 31
        cand = [
            stream_ref[base + k if k < BAND else jnp.minimum(base + k, STREAM_WORDS - 1)]
            for k in range(BAND + 2)
        ]
        for bit in (4, 2, 1):
            m = (rel & bit) != 0
            cand = [jnp.where(m, cand[k + bit], cand[k]) for k in range(bit + 2)]
        a, b, c = cand
        win = shl(a, off) | shr(shr(b, 1), 31 - off)
        nxt = shl(b, off) | shr(shr(c, 1), 31 - off)
        odd = msg_ref[9 * t + 8]
        words = []
        for h in range(2):
            g = 2 * s + h
            p0 = lax.clz(win)
            rest = win ^ shr(top, p0)
            p1 = lax.clz(rest)
            rest = rest ^ shr(top, p1)
            p2 = lax.clz(rest)
            rest = rest ^ shr(top, p2)
            p3 = lax.clz(rest)
            if h == 0:
                win = shl(shl(win, 1), p3) | shr(nxt, 31 - p3)
            pos = pos + p3 + 1
            p = p0 | shl(p1, 8) | shl(p2, 16) | shl(p3, 24)
            n = p * c32(2 - 512) - c32(0x02020200)
            n = n | ((shr(odd, 7 - g) if g < 7 else odd) & c32(0x01010101))
            ge3 = at_least(n, 3)
            d = (n ^ ((ge3 ^ c32(0x01010101)) * 3)) + ge3
            d = d + at_least(n, 10) * 9 - at_least(n, 9) * 10
            d = jnp.where(raw != 0, msg_ref[BINADES_AT + 8 * t + g], d)
            low = msg_ref[9 * t + g]
            ta = (
                (low & c32(0x007F007F))
                | (shl(low, 8) & c32(0x80008000))
                | (shl(d, 7) & c32(0x7F807F80))
            )
            tb = (
                (shr(low, 8) & c32(0x007F007F))
                | (low & c32(0x80008000))
                | (shr(d, 1) & c32(0x7F807F80))
            )
            words += [bias - ta, bias - tb]
        rows = pl.ds(pl.multiple_of(i * 32, 32) + 16 * (s // 2), 16)
        cols = pl.ds(512 * (s % 2), 512)
        out_ref[rows, cols] = pltpu.bitcast(jnp.concatenate(words, axis=1), BF16)
        return pos

    def body(i, positions):
        for s in range(4):
            positions = tuple(step(i, s, j, p) for j, p in zip(jobs, positions))
        return positions

    positions = tuple(job[2][...] for job in jobs)
    positions = lax.fori_loop(0, TICK_ITERS, body, positions)
    for job, pos in zip(jobs, positions):
        job[2][...] = pos


def all_gather_kernel(x_ref, *refs):
    outs = refs[: len(PIECE_ROWS)]
    (
        in_s, in_k, loc_s, loc_k, dec_y, dec_x,
        msg_s, msg_y, msg_x, hdr_s, hdr_y, hdr_x,
        enc_state, dec_stream, dec_pos, counter,
        in_s_sem, in_k_sem, loc_s_sem, loc_k_sem, dec_y_sem, dec_x_sem,
        y_sent, y_landed, x_sent, x_landed, y_credit, x_credit,
    ) = refs[len(PIECE_ROWS) :]

    my_x, my_y = lax.axis_index("x"), lax.axis_index("y")
    y_peer, x_peer = (my_x, 1 - my_y), (1 - my_x, my_y)
    send_row = my_x * (SHARD_ROWS // 2)
    keep_row = (1 - my_x) * (SHARD_ROWS // 2)
    own_row = my_y * SHARD_ROWS
    other_row = (1 - my_y) * SHARD_ROWS

    def load(buf, sem, row, tick):
        slot = tick % N_IN
        rows = pl.ds(pl.multiple_of(row + tick * TICK_ROWS, TICK_ROWS), TICK_ROWS)
        return pltpu.make_async_copy(x_ref.at[rows], buf.at[slot], sem.at[slot])

    def load_ahead(buf, sem, row, tick):
        @pl.when(tick + N_IN < N_TICKS)
        def _():
            load(buf, sem, row, tick + N_IN).start()

    def store(buf, sem, row, tick):
        slot = tick % N_OUT
        row = row + tick * TICK_ROWS
        start = 0
        for out, n in zip(outs, PIECE_ROWS):

            @pl.when((row >= start) & (row < start + n))
            def _(out=out, start=start):
                rows = pl.ds(pl.multiple_of(row - start, TICK_ROWS), TICK_ROWS)
                pltpu.make_async_copy(buf.at[slot], out.at[rows], sem.at[slot]).start()

            start += n

    def wait_stored(buf, sem, tick):
        slot = tick % N_OUT
        pltpu.make_async_copy(buf.at[slot], buf.at[slot], sem.at[slot]).wait()

    def copy(src, dst, peer, chunk, kind, half):
        (src_hdr, src_msg, sent), (dst_hdr, dst_msg, landed) = src, dst
        i, j = chunk % src_msg.shape[0], chunk % dst_msg.shape[0]
        if kind == HEADER:
            a, b = src_hdr.at[i], dst_hdr.at[j]
        else:
            part = {
                STREAMS: pl.ds(STREAM_AT, DENSE_WORDS + 1),
                BINADES: pl.ds(BINADES_AT, SLOT_VREGS - BINADES_AT),
                PLANES: pl.ds(half * (PLANE_VREGS // 2), PLANE_VREGS // 2),
            }[kind]
            a, b = src_msg.at[i, part], dst_msg.at[j, part]
        return pltpu.make_async_remote_copy(
            a, b, sent.at[i, kind + half], landed.at[j, kind + half],
            device_id=peer, device_id_type=MESH,
        )

    def over_y(chunk, kind, half=0):
        src, dst = (hdr_s, msg_s, y_sent), (hdr_y, msg_y, y_landed)
        return copy(src, dst, y_peer, chunk, kind, half)

    def over_x(chunk, kind, half=0):
        src, dst = (hdr_y, msg_y, x_sent), (hdr_x, msg_x, x_landed)
        return copy(src, dst, x_peer, chunk, kind, half)

    def wait_tail_sent(link, chunk, raw):
        link(chunk, HEADER).wait_send()
        link(chunk, STREAMS).wait_send()
        pl.when(raw != 0)(lambda: link(chunk, BINADES).wait_send())

    def send_own(tick):
        chunk, j = tick // TICKS, tick % TICKS
        slot = chunk % N_SEND

        @pl.when(chunk >= N_SEND)
        def _():
            old = chunk - N_SEND
            pl.when(j == 0)(lambda: wait_tail_sent(over_y, old, hdr_s[slot, 1]))
            over_y(old, PLANES, 2 * j).wait_send()
            over_y(old, PLANES, 2 * j + 1).wait_send()

        pl.when(tick >= N_OUT)(lambda: wait_stored(loc_s, loc_s_sem, tick))
        load(in_s, in_s_sem, send_row, tick).wait()

        @pl.when(tick == 0)
        def _():
            for i in range(1, N_IN):
                load(in_s, in_s_sem, send_row, i).start()
            for i in range(N_IN):
                load(in_k, in_k_sem, keep_row, i).start()

        x, msg = in_s.at[tick % N_IN], msg_s.at[slot]

        @pl.when(j == 0)
        def _():
            hdr_s[slot, 0] = encode_begin(x, msg, enc_state)

        encode_rows(x, loc_s.at[tick % N_OUT], msg, enc_state, hdr_s[slot, 0], j)
        pl.when(tick == 0)(lambda: pl.semaphore_wait(barrier, 2))
        pl.when((j == 0) & (chunk >= N_RECV))(
            lambda: pl.semaphore_wait(y_credit.at[chunk % N_RECV], 1)
        )

        @pl.when(j == TICKS - 1)
        def _():
            raw = encode_end(msg, enc_state, counter)
            hdr_s[slot, 1] = raw
            over_y(chunk, HEADER).start()
            over_y(chunk, STREAMS).start()
            pl.when(raw != 0)(lambda: over_y(chunk, BINADES).start())

        over_y(chunk, PLANES, 2 * j).start()
        over_y(chunk, PLANES, 2 * j + 1).start()
        store(loc_s, loc_s_sem, own_row + send_row, tick)
        load_ahead(in_s, in_s_sem, send_row, tick)

    def keep_own(tick):
        pl.when(tick >= N_OUT)(lambda: wait_stored(loc_k, loc_k_sem, tick))
        load(in_k, in_k_sem, keep_row, tick).wait()
        loc_k[tick % N_OUT] = in_k[tick % N_IN].astype(BF16)
        store(loc_k, loc_k_sem, own_row + keep_row, tick)
        load_ahead(in_k, in_k_sem, keep_row, tick)

    def forward(tick, h):
        chunk, j = tick // TICKS, tick % TICKS

        def relay(kind, half=0):
            over_y(chunk, kind, half).wait_recv()
            over_x(chunk, kind, half).start()

        if h == 0:
            pl.when((j == 0) & (chunk >= N_RECV))(
                lambda: pl.semaphore_wait(x_credit.at[chunk % N_RECV], 1)
            )

            @pl.when(j == TICKS - 1)
            def _():
                relay(HEADER)
                relay(STREAMS)
                pl.when(hdr_y[chunk % N_RECV, 1] != 0)(lambda: relay(BINADES))

        relay(PLANES, 2 * j + h)

    def receive(tick):
        chunk, j = tick // TICKS, tick % TICKS
        slot, o = chunk % N_RECV, tick % N_OUT

        @pl.when(j == 0)
        def _():
            over_x(chunk, HEADER).wait_recv()
            over_x(chunk, STREAMS).wait_recv()
            pl.when(hdr_x[slot, 1] != 0)(lambda: over_x(chunk, BINADES).wait_recv())
            decode_begin(msg_y.at[slot], dec_stream.at[0], dec_pos.at[0], counter)
            decode_begin(msg_x.at[slot], dec_stream.at[1], dec_pos.at[1], counter)

        over_x(chunk, PLANES, 2 * j).wait_recv()
        over_x(chunk, PLANES, 2 * j + 1).wait_recv()
        pl.when(tick >= N_OUT)(lambda: wait_stored(dec_y, dec_y_sem, tick))
        pl.when(tick >= N_OUT)(lambda: wait_stored(dec_x, dec_x_sem, tick))
        decode_rows(
            [
                (msg.at[slot], dec_stream.at[k], dec_pos.at[k], out.at[o], hdr[slot, 0], hdr[slot, 1])
                for k, (msg, hdr, out) in enumerate(((msg_y, hdr_y, dec_y), (msg_x, hdr_x, dec_x)))
            ],
            j,
        )
        store(dec_y, dec_y_sem, other_row + send_row, tick)
        store(dec_x, dec_x_sem, other_row + keep_row, tick)
        over_x(chunk, PLANES, 2 * j).wait_send()
        over_x(chunk, PLANES, 2 * j + 1).wait_send()

        @pl.when(j == TICKS - 1)
        def _():
            wait_tail_sent(over_x, chunk, hdr_y[slot, 1])

            @pl.when(chunk + N_RECV < N_CHUNKS)
            def _():
                for credit, peer in ((y_credit, y_peer), (x_credit, x_peer)):
                    pl.semaphore_signal(credit.at[slot], inc=1, device_id=peer, device_id_type=MESH)

    barrier = pltpu.get_barrier_semaphore()
    load(in_s, in_s_sem, send_row, 0).start()
    for peer in (y_peer, x_peer):
        pl.semaphore_signal(barrier, inc=1, device_id=peer, device_id_type=MESH)
    r = lax.broadcasted_iota(I32, (128, 256), 0)
    q = lax.broadcasted_iota(I32, (128, 256), 1)
    counter[...] = jnp.where(r < q, 1.0, 0.0).astype(BF16)

    def run_tick(tick, _):
        relayed = tick - FORWARD_LAG
        relaying = (tick >= FORWARD_LAG) & (tick < N_TICKS + FORWARD_LAG)
        pl.when(tick < N_TICKS)(lambda: send_own(tick))
        pl.when(relaying)(lambda: forward(relayed, 0))
        pl.when(tick < N_TICKS)(lambda: keep_own(tick))
        pl.when(tick >= DECODE_LAG)(lambda: receive(tick - DECODE_LAG))
        pl.when(relaying)(lambda: forward(relayed, 1))

    lax.fori_loop(0, N_TICKS + DECODE_LAG, run_tick, None)

    for chunk in range(N_CHUNKS - N_SEND, N_CHUNKS):
        wait_tail_sent(over_y, chunk, hdr_s[chunk % N_SEND, 1])
        for half in range(2 * TICKS):
            over_y(chunk, PLANES, half).wait_send()
    for tick in range(N_TICKS - N_OUT, N_TICKS):
        wait_stored(loc_s, loc_s_sem, tick)
        wait_stored(loc_k, loc_k_sem, tick)
        wait_stored(dec_y, dec_y_sem, tick)
        wait_stored(dec_x, dec_x_sem, tick)


def pallas_dist_ag_xy_y_m65536_n1024_kernel(x: jax.Array):
    assert x.shape == (SHARD_ROWS, COLS) and x.dtype == jnp.float32
    dma = pltpu.SemaphoreType.DMA
    n_copies = PLANES + 2 * TICKS
    *pieces, rest = pl.pallas_call(
        all_gather_kernel,
        out_shape=(
            *[pltpu.VMEM((n, COLS), BF16) for n in PIECE_ROWS[:-1]],
            jax.ShapeDtypeStruct((PIECE_ROWS[-1], COLS), BF16),
        ),
        in_specs=[pl.BlockSpec(memory_space=pl.ANY)],
        out_specs=(
            *[pl.BlockSpec(memory_space=pltpu.VMEM) for _ in PIECE_ROWS[:-1]],
            pl.BlockSpec(memory_space=pl.ANY),
        ),
        scratch_shapes=[
            *[pltpu.VMEM((N_IN, TICK_ROWS, COLS), jnp.float32)] * 2,
            *[pltpu.VMEM((N_OUT, TICK_ROWS, COLS), BF16)] * 4,
            *[pltpu.VMEM((n, SLOT_VREGS, 8, 128), I32) for n in (N_SEND, N_RECV, N_RECV)],
            *[pltpu.SMEM((n, 2), I32) for n in (N_SEND, N_RECV, N_RECV)],
            pltpu.VMEM((5, 8, 128), I32),
            pltpu.VMEM((2, STREAM_WORDS, 8, 128), I32),
            pltpu.VMEM((2, 8, 128), I32),
            pltpu.VMEM((128, 256), BF16),
            *[dma((N_IN,))] * 2,
            *[dma((N_OUT,))] * 4,
            *[dma((n, n_copies)) for n in (N_SEND, N_RECV, N_RECV, N_RECV)],
            *[pltpu.SemaphoreType.REGULAR((N_RECV,))] * 2,
        ],
        compiler_params=pltpu.CompilerParams(collective_id=0),
    )(x)
    start = 0
    for n in STAGED_TICKS:
        pieces.append(lax.optimization_barrier(rest[start : start + n * TICK_ROWS]))
        start += n * TICK_ROWS
    return jnp.concatenate([*pieces, rest[start:]], axis=0)
```

```python
import functools

import jax
import jax.numpy as jnp
import numpy as np
from jax import lax
from jax.experimental import pallas as pl
from jax.experimental.pallas import tpu as pltpu

SHARD_ROWS = 65536
COLS = 1024

TICK_ROWS = 128
TICKS = 4
STREAM_WORDS = 30
DENSE_WORDS = 26
BAND = 8
TOP_OFFSET = 456

FORWARD_LAG = 2
DECODE_LAG = 6
N_IN = 2
N_OUT = 2
N_SEND = 2
N_RECV = 3
VMEM_TICKS = (447, 1)
STAGED_TICKS = (281, 293)

CHUNK_ROWS = TICKS * TICK_ROWS
N_TICKS = SHARD_ROWS // 2 // TICK_ROWS
N_CHUNKS = N_TICKS // TICKS
TICK_ITERS = TICK_ROWS // 32
PLANE_VREGS = 9 * TICK_ITERS
STREAM_AT = TICKS * PLANE_VREGS
BINADES_AT = STREAM_AT + STREAM_WORDS
BINADE_VREGS = 8 * TICK_ITERS
SLOT_VREGS = BINADES_AT + TICKS * BINADE_VREGS
RESULT_TICKS = (*VMEM_TICKS, 4 * N_TICKS - sum(VMEM_TICKS))

I32 = jnp.int32
BF16 = jnp.bfloat16
MESH = pl.DeviceIdType.MESH
HEADER, PLANES, STREAMS, BINADES = range(4)
LANDED_SEM = (0, 1, 1 + 2 * TICKS, 1 + 2 * TICKS)
shr = lax.shift_right_logical
shl = lax.shift_left


def c32(v):
    return np.uint32(v & 0xFFFFFFFF).astype(np.int32)


def at_least(x, k):
    return shr(x + c32(0x01010101 * (128 - k)), 7) & c32(0x01010101)


def band_base(group):
    typical = shr(group * 209 + 768, 10)
    return jnp.clip(typical - BAND // 2, 0, STREAM_WORDS - BAND)


def lane_counts(flags, counter_ref):
    ones = jnp.where(flags, 1.0, 0.0).astype(BF16)
    counts = jnp.dot(ones, counter_ref[...], preferred_element_type=jnp.float32)
    counts = counts.astype(I32)
    return counts[:, :128], counts[:, 128:]


def store_word(msg_ref, base, word_idx, word):
    rel = word_idx - base
    for i in range(BAND):
        pltpu.store(msg_ref.at[STREAM_AT + base + i], word, mask=rel == i)
    return shr(rel, 3)


def encode_begin(x_ref, msg_ref, state_ref):
    w = pltpu.bitcast(x_ref[0:16, :].astype(BF16), I32)
    mean_magnitude = shr(jnp.sum((w & 0x7FFF) + (shr(w, 16) & 0x7FFF)), 14)
    zero = jnp.zeros((8, 128), I32)
    for i in range(STREAM_WORDS):
        msg_ref[STREAM_AT + i] = zero
    for i in range(state_ref.shape[0]):
        state_ref[i] = zero
    return (mean_magnitude + TOP_OFFSET + 0x8000) * 0x10001


def encode_rows(x_ref, loc_ref, msg_ref, state_ref, bias, tick):
    top = jnp.full((8, 128), c32(0x80000000), I32)

    def body(i, carry):
        acc, off, word_idx, bad, binades = carry
        t = tick * TICK_ITERS + i
        odd = None
        for s in range(4):
            rows = pl.ds(pl.multiple_of(i * 32, 32) + 16 * (s // 2), 16)
            cols = pl.ds(512 * (s % 2), 512)
            b = x_ref[rows, cols].astype(BF16)
            loc_ref[rows, cols] = b
            w = bias - pltpu.bitcast(b, I32)
            for h in range(2):
                g = 2 * s + h
                ta = w[:, 256 * h : 256 * h + 128]
                tb = w[:, 256 * h + 128 : 256 * h + 256]
                msg_ref[9 * t + g] = (
                    (ta & c32(0x007F007F))
                    | (shr(ta, 8) & c32(0x00800080))
                    | (shl(tb, 8) & c32(0x7F007F00))
                    | (tb & c32(0x80008000))
                )
                d = (shr(ta, 7) & c32(0x00FF00FF)) | (shl(tb, 1) & c32(0xFF00FF00))
                msg_ref[BINADES_AT + 8 * t + g] = d
                binades = binades | d
                ge4 = at_least(d, 4)
                n = (d ^ ((ge4 ^ c32(0x01010101)) * 3)) - ge4 + at_least(d, 10)
                n = n + c32(0x06060606) - at_least(d, 1) * 6
                last = n & c32(0x01010101)
                odd = last if odd is None else (shl(odd, 1) | last)
                p = (shr(n, 1) & c32(0x1F1F1F1F)) + c32(0x01010100)
                p = p * c32(0x01010101)
                p3 = shr(p, 24)
                bad = bad | shr(p3, 5)
                p3 = p3 & 31
                code = (
                    shr(top, p & 31)
                    | shr(top, shr(p, 8) & 31)
                    | shr(top, shr(p, 16) & 31)
                    | shr(top, p3)
                )
                word = acc | shr(code, off)
                bad = bad | store_word(msg_ref, band_base(8 * t + g), word_idx, word)
                end = off + p3 + 1
                full = shr(end, 5)
                acc = jnp.where(full != 0, shl(shl(code, 1), 31 - off), word)
                off = end & 31
                word_idx = word_idx + full
        msg_ref[9 * t + 8] = odd
        return acc, off, word_idx, bad, binades

    state = tuple(state_ref[i] for i in range(state_ref.shape[0]))
    state = lax.fori_loop(0, TICK_ITERS, body, state)
    for i, value in enumerate(state):
        state_ref[i] = value


def encode_end(msg_ref, state_ref, counter_ref):
    acc, off, word_idx, bad, binades = (state_ref[i] for i in range(5))
    lost = store_word(msg_ref, STREAM_WORDS - BAND, word_idx, acc)
    bad = bad | jnp.where(off != 0, lost, 0) | (binades & c32(0xC0C0C0C0))

    n_words = word_idx + jnp.where(off != 0, 1, 0)
    pooled = range(DENSE_WORDS, STREAM_WORDS)
    used = jnp.concatenate([n_words > i for i in pooled], axis=0)
    before, total = lane_counts(used, counter_ref)
    lane = lax.broadcasted_iota(I32, used.shape, 1)
    val = jnp.concatenate([msg_ref[STREAM_AT + i] for i in pooled], axis=0)
    move = jnp.where(used, lane - before, 0)
    for k in (1, 2, 4, 8, 16, 32, 64):
        val_in, move_in = pltpu.roll(val, 128 - k, 1), pltpu.roll(move, 128 - k, 1)
        take = (move_in & k) != 0
        val = jnp.where(take, val_in, val)
        move = jnp.where(take, move_in, jnp.where((move & k) != 0, 0, move))
    pool, filled = val[0:8], total[0:8]
    for i in range(1, len(pooled)):
        slot = lane[0:8] - filled
        more = jnp.take_along_axis(val[8 * i : 8 * i + 8], slot & 127, axis=1)
        pool = jnp.where(slot < 0, pool, more)
        filled = filled + total[8 * i : 8 * i + 8]
    msg_ref[STREAM_AT + DENSE_WORDS] = pool
    bad = bad | jnp.where(filled > 128, 1, 0)
    return jnp.max(jnp.where(bad != 0, 1, 0))


def decode_begin(msg_ref, stream_ref, pos_ref, counter_ref):
    markers = []
    for i in range(DENSE_WORDS):
        word = msg_ref[STREAM_AT + i]
        stream_ref[i] = word
        markers.append(lax.population_count(word))
    markers = functools.reduce(jnp.add, markers)
    pool, filled = msg_ref[STREAM_AT + DENSE_WORDS], 0
    for i in range(DENSE_WORDS, STREAM_WORDS):
        used = markers < CHUNK_ROWS
        before, total = lane_counts(used, counter_ref)
        word = jnp.take_along_axis(pool, (filled + before) & 127, axis=1)
        word = jnp.where(used, word, 0)
        stream_ref[i] = word
        markers = markers + lax.population_count(word)
        filled = filled + total
    pos_ref[...] = jnp.zeros((8, 128), I32)


def decode_rows(jobs, tick):
    top = jnp.full((8, 128), c32(0x80000000), I32)

    def step(i, s, job, pos):
        msg_ref, stream_ref, _, out_ref, bias, raw = job
        t = tick * TICK_ITERS + i
        base = band_base(8 * t + 2 * s)
        rel = shr(pos, 5) - base
        off = pos & 31
        cand = [
            stream_ref[base + k if k < BAND else jnp.minimum(base + k, STREAM_WORDS - 1)]
            for k in range(BAND + 2)
        ]
        for bit in (4, 2, 1):
            m = (rel & bit) != 0
            cand = [jnp.where(m, cand[k + bit], cand[k]) for k in range(bit + 2)]
        a, b, c = cand
        win = shl(a, off) | shr(shr(b, 1), 31 - off)
        nxt = shl(b, off) | shr(shr(c, 1), 31 - off)
        odd = msg_ref[9 * t + 8]
        words = []
        for h in range(2):
            g = 2 * s + h
            p0 = lax.clz(win)
            rest = win ^ shr(top, p0)
            p1 = lax.clz(rest)
            rest = rest ^ shr(top, p1)
            p2 = lax.clz(rest)
            rest = rest ^ shr(top, p2)
            p3 = lax.clz(rest)
            if h == 0:
                win = shl(shl(win, 1), p3) | shr(nxt, 31 - p3)
            pos = pos + p3 + 1
            p = p0 | shl(p1, 8) | shl(p2, 16) | shl(p3, 24)
            n = p * c32(2 - 512) - c32(0x02020200)
            n = n | ((shr(odd, 7 - g) if g < 7 else odd) & c32(0x01010101))
            ge3 = at_least(n, 3)
            d = (n ^ ((ge3 ^ c32(0x01010101)) * 3)) + ge3
            d = d + at_least(n, 10) * 9 - at_least(n, 9) * 10
            d = jnp.where(raw != 0, msg_ref[BINADES_AT + 8 * t + g], d)
            low = msg_ref[9 * t + g]
            ta = (
                (low & c32(0x007F007F))
                | (shl(low, 8) & c32(0x80008000))
                | (shl(d, 7) & c32(0x7F807F80))
            )
            tb = (
                (shr(low, 8) & c32(0x007F007F))
                | (low & c32(0x80008000))
                | (shr(d, 1) & c32(0x7F807F80))
            )
            words += [bias - ta, bias - tb]
        rows = pl.ds(pl.multiple_of(i * 32, 32) + 16 * (s // 2), 16)
        cols = pl.ds(512 * (s % 2), 512)
        out_ref[rows, cols] = pltpu.bitcast(jnp.concatenate(words, axis=1), BF16)
        return pos

    def body(i, positions):
        for s in range(4):
            positions = tuple(step(i, s, j, p) for j, p in zip(jobs, positions))
        return positions

    positions = tuple(job[2][...] for job in jobs)
    positions = lax.fori_loop(0, TICK_ITERS, body, positions)
    for job, pos in zip(jobs, positions):
        job[2][...] = pos


def all_gather_kernel(x_ref, *refs):
    outs = refs[: len(RESULT_TICKS)]
    (
        in_s, in_k, loc_s, loc_k, dec_y, dec_x,
        msg_s, msg_y, msg_x, hdr_s, hdr_y, hdr_x,
        enc_state, dec_stream, dec_pos, counter,
        in_s_sem, in_k_sem, loc_s_sem, loc_k_sem, dec_y_sem, dec_x_sem,
        y_sent, y_landed, x_sent, x_landed, y_credit, x_credit,
    ) = refs[len(RESULT_TICKS) :]

    my_x, my_y = lax.axis_index("x"), lax.axis_index("y")
    y_peer, x_peer = (my_x, 1 - my_y), (1 - my_x, my_y)
    send_at = my_x * N_TICKS
    keep_at = (1 - my_x) * N_TICKS
    own_at = my_y * 2 * N_TICKS
    other_at = (1 - my_y) * 2 * N_TICKS

    def load(buf, sem, at, tick):
        slot = tick % N_IN
        rows = pl.ds(pl.multiple_of((at + tick) * TICK_ROWS, TICK_ROWS), TICK_ROWS)
        return pltpu.make_async_copy(x_ref.at[rows], buf.at[slot], sem.at[slot])

    def load_ahead(buf, sem, at, tick):
        @pl.when(tick + N_IN < N_TICKS)
        def _():
            load(buf, sem, at, tick + N_IN).start()

    def store(buf, sem, at, tick):
        slot = tick % N_OUT
        at = at + tick
        for out in outs:

            @pl.when((at >= 0) & (at < out.shape[0]))
            def _(out=out, at=at):
                pltpu.make_async_copy(buf.at[slot], out.at[at], sem.at[slot]).start()

            at = at - out.shape[0]

    def wait_stored(buf, sem, tick):
        slot = tick % N_OUT
        pltpu.make_async_copy(buf.at[slot], buf.at[slot], sem.at[slot]).wait()

    def copy(src, dst, peer, chunk, kind, part):
        (src_hdr, src_msg, sent), (dst_hdr, dst_msg, landed) = src, dst
        i, j = chunk % src_msg.shape[0], chunk % dst_msg.shape[0]
        if kind == HEADER:
            a, b = src_hdr.at[i], dst_hdr.at[j]
        else:
            vregs = {
                PLANES: pl.ds(part * (PLANE_VREGS // 2), PLANE_VREGS // 2),
                STREAMS: pl.ds(STREAM_AT, DENSE_WORDS + 1),
                BINADES: pl.ds(BINADES_AT + part * BINADE_VREGS, BINADE_VREGS),
            }[kind]
            a, b = src_msg.at[i, vregs], dst_msg.at[j, vregs]
        sent_sem = sent.at[i, min(kind, STREAMS)]
        landed_sem = landed.at[j, LANDED_SEM[kind] + part]
        return pltpu.make_async_remote_copy(
            a, b, sent_sem, landed_sem, device_id=peer, device_id_type=MESH
        )

    def over_y(chunk, kind, part=0):
        src, dst = (hdr_s, msg_s, y_sent), (hdr_y, msg_y, y_landed)
        return copy(src, dst, y_peer, chunk, kind, part)

    def over_x(chunk, kind, part=0):
        src, dst = (hdr_y, msg_y, x_sent), (hdr_x, msg_x, x_landed)
        return copy(src, dst, x_peer, chunk, kind, part)

    def with_tail(raw, action):
        pl.when(raw == 0)(lambda: action(STREAMS, 0))

        @pl.when(raw != 0)
        def _():
            for part in range(TICKS):
                action(BINADES, part)

    def wait_sent(link, msg, sent, chunk, raw):
        slot = chunk % msg.shape[0]
        planes = msg.at[slot, pl.ds(0, STREAM_AT)]
        link(chunk, HEADER).wait_send()
        pltpu.make_async_copy(planes, planes, sent.at[slot, PLANES]).wait()
        with_tail(raw, lambda kind, part: link(chunk, kind, part).wait_send())

    def send_own(tick):
        chunk, j = tick // TICKS, tick % TICKS
        slot = chunk % N_SEND

        @pl.when((j == 0) & (chunk >= N_SEND))
        def _():
            wait_sent(over_y, msg_s, y_sent, chunk - N_SEND, hdr_s[slot, 1])

        pl.when(tick >= N_OUT)(lambda: wait_stored(loc_s, loc_s_sem, tick))
        load(in_s, in_s_sem, send_at, tick).wait()

        @pl.when(tick == 0)
        def _():
            for i in range(1, N_IN):
                load(in_s, in_s_sem, send_at, i).start()
            for i in range(N_IN):
                load(in_k, in_k_sem, keep_at, i).start()

        x, msg = in_s.at[tick % N_IN], msg_s.at[slot]

        @pl.when(j == 0)
        def _():
            hdr_s[slot, 0] = encode_begin(x, msg, enc_state)

        encode_rows(x, loc_s.at[tick % N_OUT], msg, enc_state, hdr_s[slot, 0], j)
        pl.when(tick == 0)(lambda: pl.semaphore_wait(barrier, 2))
        pl.when((j == 0) & (chunk >= N_RECV))(
            lambda: pl.semaphore_wait(y_credit.at[chunk % N_RECV], 1)
        )

        @pl.when(j == TICKS - 1)
        def _():
            raw = encode_end(msg, enc_state, counter)
            hdr_s[slot, 1] = raw
            over_y(chunk, HEADER).start()
            with_tail(raw, lambda kind, part: over_y(chunk, kind, part).start())

        over_y(chunk, PLANES, 2 * j).start()
        over_y(chunk, PLANES, 2 * j + 1).start()
        store(loc_s, loc_s_sem, own_at + send_at, tick)
        load_ahead(in_s, in_s_sem, send_at, tick)

    def keep_own(tick):
        pl.when(tick >= N_OUT)(lambda: wait_stored(loc_k, loc_k_sem, tick))
        load(in_k, in_k_sem, keep_at, tick).wait()
        loc_k[tick % N_OUT] = in_k[tick % N_IN].astype(BF16)
        store(loc_k, loc_k_sem, own_at + keep_at, tick)
        load_ahead(in_k, in_k_sem, keep_at, tick)

    def forward(tick, h):
        chunk, j = tick // TICKS, tick % TICKS

        def relay(kind, part=0):
            over_y(chunk, kind, part).wait_recv()
            over_x(chunk, kind, part).start()

        if h == 0:
            pl.when((j == 0) & (chunk >= N_RECV))(
                lambda: pl.semaphore_wait(x_credit.at[chunk % N_RECV], 1)
            )

            @pl.when(j == TICKS - 1)
            def _():
                relay(HEADER)
                with_tail(hdr_y[chunk % N_RECV, 1], relay)

        relay(PLANES, 2 * j + h)

    def receive(tick):
        chunk, j = tick // TICKS, tick % TICKS
        slot, o = chunk % N_RECV, tick % N_OUT

        @pl.when(j == 0)
        def _():
            over_x(chunk, HEADER).wait_recv()
            with_tail(
                hdr_x[slot, 1], lambda kind, part: over_x(chunk, kind, part).wait_recv()
            )
            decode_begin(msg_y.at[slot], dec_stream.at[0], dec_pos.at[0], counter)
            decode_begin(msg_x.at[slot], dec_stream.at[1], dec_pos.at[1], counter)

        over_x(chunk, PLANES, 2 * j).wait_recv()
        over_x(chunk, PLANES, 2 * j + 1).wait_recv()
        pl.when(tick >= N_OUT)(lambda: wait_stored(dec_y, dec_y_sem, tick))
        pl.when(tick >= N_OUT)(lambda: wait_stored(dec_x, dec_x_sem, tick))
        decode_rows(
            [
                (msg.at[slot], dec_stream.at[k], dec_pos.at[k], out.at[o], hdr[slot, 0], hdr[slot, 1])
                for k, (msg, hdr, out) in enumerate(((msg_y, hdr_y, dec_y), (msg_x, hdr_x, dec_x)))
            ],
            j,
        )
        store(dec_y, dec_y_sem, other_at + send_at, tick)
        store(dec_x, dec_x_sem, other_at + keep_at, tick)

        @pl.when(j == TICKS - 1)
        def _():
            wait_sent(over_x, msg_y, x_sent, chunk, hdr_y[slot, 1])

            @pl.when(chunk + N_RECV < N_CHUNKS)
            def _():
                for credit, peer in ((y_credit, y_peer), (x_credit, x_peer)):
                    pl.semaphore_signal(credit.at[slot], inc=1, device_id=peer, device_id_type=MESH)

    barrier = pltpu.get_barrier_semaphore()
    load(in_s, in_s_sem, send_at, 0).start()

    def clear_tails(i, _):
        for msg in (msg_y, msg_x):
            for slot in range(N_RECV):
                msg[slot, i] = jnp.zeros((8, 128), I32)

    lax.fori_loop(STREAM_AT, SLOT_VREGS, clear_tails, None)
    for peer in (y_peer, x_peer):
        pl.semaphore_signal(barrier, inc=1, device_id=peer, device_id_type=MESH)
    r = lax.broadcasted_iota(I32, (128, 256), 0)
    q = lax.broadcasted_iota(I32, (128, 256), 1)
    counter[...] = jnp.where(r < q, 1.0, 0.0).astype(BF16)

    def run_tick(tick, _):
        relayed = tick - FORWARD_LAG
        relaying = (tick >= FORWARD_LAG) & (tick < N_TICKS + FORWARD_LAG)
        pl.when(tick < N_TICKS)(lambda: send_own(tick))
        pl.when(relaying)(lambda: forward(relayed, 0))
        pl.when(tick < N_TICKS)(lambda: keep_own(tick))
        pl.when(tick >= DECODE_LAG)(lambda: receive(tick - DECODE_LAG))
        pl.when(relaying)(lambda: forward(relayed, 1))

    lax.fori_loop(0, N_TICKS + DECODE_LAG, run_tick, None)

    for chunk in range(N_CHUNKS - N_SEND, N_CHUNKS):
        wait_sent(over_y, msg_s, y_sent, chunk, hdr_s[chunk % N_SEND, 1])
    for tick in range(N_TICKS - N_OUT, N_TICKS):
        wait_stored(loc_s, loc_s_sem, tick)
        wait_stored(loc_k, loc_k_sem, tick)
        wait_stored(dec_y, dec_y_sem, tick)
        wait_stored(dec_x, dec_x_sem, tick)


def pallas_dist_ag_xy_y_m65536_n1024_kernel(x: jax.Array):
    assert x.shape == (SHARD_ROWS, COLS) and x.dtype == jnp.float32
    dma = pltpu.SemaphoreType.DMA
    n_copies = 1 + 3 * TICKS
    *pieces, rest = pl.pallas_call(
        all_gather_kernel,
        out_shape=(
            *[pltpu.VMEM((n, TICK_ROWS, COLS), BF16) for n in VMEM_TICKS],
            jax.ShapeDtypeStruct((RESULT_TICKS[-1], TICK_ROWS, COLS), BF16),
        ),
        in_specs=[pl.BlockSpec(memory_space=pl.ANY)],
        out_specs=(
            *[pl.BlockSpec(memory_space=pltpu.VMEM) for _ in VMEM_TICKS],
            pl.BlockSpec(memory_space=pl.ANY),
        ),
        scratch_shapes=[
            *[pltpu.VMEM((N_IN, TICK_ROWS, COLS), jnp.float32)] * 2,
            *[pltpu.VMEM((N_OUT, TICK_ROWS, COLS), BF16)] * 4,
            *[pltpu.VMEM((n, SLOT_VREGS, 8, 128), I32) for n in (N_SEND, N_RECV, N_RECV)],
            *[pltpu.SMEM((n, 2), I32) for n in (N_SEND, N_RECV, N_RECV)],
            pltpu.VMEM((5, 8, 128), I32),
            pltpu.VMEM((2, STREAM_WORDS, 8, 128), I32),
            pltpu.VMEM((2, 8, 128), I32),
            pltpu.VMEM((128, 256), BF16),
            *[dma((N_IN,))] * 2,
            *[dma((N_OUT,))] * 4,
            dma((N_SEND, 3)),
            dma((N_RECV, n_copies)),
            dma((N_RECV, 3)),
            dma((N_RECV, n_copies)),
            *[pltpu.SemaphoreType.REGULAR((N_RECV,))] * 2,
        ],
        compiler_params=pltpu.CompilerParams(collective_id=0),
    )(x)
    start = 0
    for n in STAGED_TICKS:
        pieces.append(lax.optimization_barrier(rest[start : start + n]))
        start += n
    return jnp.concatenate([*pieces, rest[start:]]).reshape(2 * SHARD_ROWS, COLS)
```

```python
import functools

import jax
import jax.numpy as jnp
import numpy as np
from jax import lax
from jax.experimental import pallas as pl
from jax.experimental.pallas import tpu as pltpu

SHARD_ROWS = 65536
COLS = 1024

TICK_ROWS = 128
TICKS = 4
STREAM_WORDS = 30
DENSE_WORDS = 26
BAND = 8
TOP_OFFSET = 456

RELAY_LAG = 2
DECODE_LAG = 6
N_IN = 2
N_OUT = 2
N_SEND = 2
N_RECV = 3

VMEM_TICKS = (447, 1)
STAGED_TICKS = (281, 293)

CHUNK_ROWS = TICKS * TICK_ROWS
N_TICKS = SHARD_ROWS // 2 // TICK_ROWS
N_CHUNKS = N_TICKS // TICKS
TICK_ITERS = TICK_ROWS // 32
HBM_TICKS = 4 * N_TICKS - sum(VMEM_TICKS)

PLANE_VREGS = 9 * TICK_ITERS
BINADE_VREGS = 8 * TICK_ITERS
STREAM_AT = TICKS * PLANE_VREGS
BINADES_AT = STREAM_AT + STREAM_WORDS
SLOT_VREGS = BINADES_AT + TICKS * BINADE_VREGS

HEADER, PLANES, STREAMS, BINADES = range(4)
FIRST_LANDED_SEM = (0, 1, 1 + 2 * TICKS, 1 + 2 * TICKS)

I32 = jnp.int32
BF16 = jnp.bfloat16
MESH = pl.DeviceIdType.MESH
shr = lax.shift_right_logical
shl = lax.shift_left


def c32(bits):
    return np.uint32(bits & 0xFFFFFFFF).astype(np.int32)


ONES = c32(0x01010101)


def at_least(x, k):
    return shr(x + c32(0x01010101 * (128 - k)), 7) & ONES


def band_base(group):
    typical = shr(group * 209 + 768, 10)
    return jnp.clip(typical - BAND // 2, 0, STREAM_WORDS - BAND)


def lane_counts(flags, counter_ref):
    ones = jnp.where(flags, 1.0, 0.0).astype(BF16)
    counts = jnp.dot(ones, counter_ref[...], preferred_element_type=jnp.float32)
    counts = counts.astype(I32)
    return counts[:, :128], counts[:, 128:]


def block(i, s):
    rows = pl.ds(pl.multiple_of(i * 32, 32) + 16 * (s // 2), 16)
    return rows, pl.ds(512 * (s % 2), 512)


def store_word(msg_ref, base, word_idx, word):
    rel = word_idx - base
    for i in range(BAND):
        pltpu.store(msg_ref.at[STREAM_AT + base + i], word, mask=rel == i)
    return shr(rel, 3)


def encode_begin(x_ref, msg_ref, state_ref):
    w = pltpu.bitcast(x_ref[0:16, :].astype(BF16), I32)
    mean_magnitude = shr(jnp.sum((w & 0x7FFF) + (shr(w, 16) & 0x7FFF)), 14)
    zero = jnp.zeros((8, 128), I32)
    for i in range(STREAM_WORDS):
        msg_ref[STREAM_AT + i] = zero
    for i in range(state_ref.shape[0]):
        state_ref[i] = zero
    return (mean_magnitude + TOP_OFFSET + 0x8000) * 0x10001


def encode_rows(x_ref, loc_ref, msg_ref, state_ref, bias, tick):
    top = jnp.full((8, 128), c32(0x80000000), I32)

    def body(i, carry):
        acc, off, word_idx, bad, binades = carry
        t = tick * TICK_ITERS + i
        odd = None
        for s in range(4):
            b = x_ref[block(i, s)].astype(BF16)
            loc_ref[block(i, s)] = b
            w = bias - pltpu.bitcast(b, I32)
            for h in range(2):
                g = 2 * s + h
                ta = w[:, 256 * h : 256 * h + 128]
                tb = w[:, 256 * h + 128 : 256 * h + 256]
                msg_ref[9 * t + g] = (
                    (ta & c32(0x007F007F))
                    | (shr(ta, 8) & c32(0x00800080))
                    | (shl(tb, 8) & c32(0x7F007F00))
                    | (tb & c32(0x80008000))
                )
                d = (shr(ta, 7) & c32(0x00FF00FF)) | (shl(tb, 1) & c32(0xFF00FF00))
                msg_ref[BINADES_AT + 8 * t + g] = d
                binades = binades | d
                ge4 = at_least(d, 4)
                n = (d ^ ((ge4 ^ ONES) * 3)) - ge4 + at_least(d, 10)
                n = n + c32(0x06060606) - at_least(d, 1) * 6
                odd = n & ONES if odd is None else shl(odd, 1) | (n & ONES)
                p = ((shr(n, 1) & c32(0x1F1F1F1F)) + c32(0x01010100)) * ONES
                last = shr(p, 24)
                bad = bad | shr(last, 5)
                last = last & 31
                code = (
                    shr(top, p & 31)
                    | shr(top, shr(p, 8) & 31)
                    | shr(top, shr(p, 16) & 31)
                    | shr(top, last)
                )
                word = acc | shr(code, off)
                bad = bad | store_word(msg_ref, band_base(8 * t + g), word_idx, word)
                end = off + last + 1
                full = shr(end, 5)
                acc = jnp.where(full != 0, shl(shl(code, 1), 31 - off), word)
                off = end & 31
                word_idx = word_idx + full
        msg_ref[9 * t + 8] = odd
        return acc, off, word_idx, bad, binades

    state = tuple(state_ref[i] for i in range(state_ref.shape[0]))
    state = lax.fori_loop(0, TICK_ITERS, body, state)
    for i, value in enumerate(state):
        state_ref[i] = value


def encode_end(msg_ref, state_ref, counter_ref):
    acc, off, word_idx, bad, binades = (state_ref[i] for i in range(5))
    lost = store_word(msg_ref, STREAM_WORDS - BAND, word_idx, acc)
    bad = bad | jnp.where(off != 0, lost, 0) | (binades & c32(0xC0C0C0C0))

    n_words = word_idx + jnp.where(off != 0, 1, 0)
    pooled = range(DENSE_WORDS, STREAM_WORDS)
    used = jnp.concatenate([n_words > i for i in pooled], axis=0)
    before, total = lane_counts(used, counter_ref)
    lane = lax.broadcasted_iota(I32, used.shape, 1)
    val = jnp.concatenate([msg_ref[STREAM_AT + i] for i in pooled], axis=0)
    move = jnp.where(used, lane - before, 0)
    for k in (1, 2, 4, 8, 16, 32, 64):
        val_in, move_in = pltpu.roll(val, 128 - k, 1), pltpu.roll(move, 128 - k, 1)
        take = (move_in & k) != 0
        val = jnp.where(take, val_in, val)
        move = jnp.where(take, move_in, jnp.where((move & k) != 0, 0, move))
    pool, filled = val[0:8], total[0:8]
    for i in range(1, len(pooled)):
        slot = lane[0:8] - filled
        more = jnp.take_along_axis(val[8 * i : 8 * i + 8], slot & 127, axis=1)
        pool = jnp.where(slot < 0, pool, more)
        filled = filled + total[8 * i : 8 * i + 8]
    msg_ref[STREAM_AT + DENSE_WORDS] = pool
    bad = bad | jnp.where(filled > 128, 1, 0)
    return jnp.max(jnp.where(bad != 0, 1, 0))


def decode_begin(msg_ref, stream_ref, pos_ref, counter_ref):
    seen = []
    for i in range(DENSE_WORDS):
        word = msg_ref[STREAM_AT + i]
        stream_ref[i] = word
        seen.append(lax.population_count(word))
    seen = functools.reduce(jnp.add, seen)
    pool, filled = msg_ref[STREAM_AT + DENSE_WORDS], 0
    for i in range(DENSE_WORDS, STREAM_WORDS):
        used = seen < CHUNK_ROWS
        before, total = lane_counts(used, counter_ref)
        word = jnp.take_along_axis(pool, (filled + before) & 127, axis=1)
        word = jnp.where(used, word, 0)
        stream_ref[i] = word
        seen = seen + lax.population_count(word)
        filled = filled + total
    pos_ref[...] = jnp.zeros((8, 128), I32)


def decode_rows(jobs, tick):
    top = jnp.full((8, 128), c32(0x80000000), I32)

    def step(i, s, job, pos):
        msg_ref, stream_ref, _, out_ref, bias, raw = job
        t = tick * TICK_ITERS + i
        base = band_base(8 * t + 2 * s)
        rel, off = shr(pos, 5) - base, pos & 31
        near = [stream_ref[base + k] for k in range(BAND)] + [
            stream_ref[jnp.minimum(base + k, STREAM_WORDS - 1)]
            for k in (BAND, BAND + 1)
        ]
        for bit in (4, 2, 1):
            up = (rel & bit) != 0
            near = [jnp.where(up, near[k + bit], near[k]) for k in range(bit + 2)]
        bits = shl(near[0], off) | shr(shr(near[1], 1), 31 - off)
        later = shl(near[1], off) | shr(shr(near[2], 1), 31 - off)
        odd = msg_ref[9 * t + 8]
        words = []
        for h in range(2):
            g = 2 * s + h
            p0 = lax.clz(bits)
            rest = bits ^ shr(top, p0)
            p1 = lax.clz(rest)
            rest = rest ^ shr(top, p1)
            p2 = lax.clz(rest)
            rest = rest ^ shr(top, p2)
            p3 = lax.clz(rest)
            if h == 0:
                bits = shl(shl(bits, 1), p3) | shr(later, 31 - p3)
            pos = pos + p3 + 1
            p = p0 | shl(p1, 8) | shl(p2, 16) | shl(p3, 24)
            n = p * c32(2 - 512) - c32(0x02020200)
            n = n | ((shr(odd, 7 - g) if g < 7 else odd) & ONES)
            ge3 = at_least(n, 3)
            d = (n ^ ((ge3 ^ ONES) * 3)) + ge3
            d = d + at_least(n, 10) * 9 - at_least(n, 9) * 10
            d = jnp.where(raw != 0, msg_ref[BINADES_AT + 8 * t + g], d)
            low = msg_ref[9 * t + g]
            ta = (
                (low & c32(0x007F007F))
                | (shl(low, 8) & c32(0x80008000))
                | (shl(d, 7) & c32(0x7F807F80))
            )
            tb = (
                (shr(low, 8) & c32(0x007F007F))
                | (low & c32(0x80008000))
                | (shr(d, 1) & c32(0x7F807F80))
            )
            words += [bias - ta, bias - tb]
        out_ref[block(i, s)] = pltpu.bitcast(jnp.concatenate(words, axis=1), BF16)
        return pos

    def body(i, positions):
        for s in range(4):
            positions = tuple(step(i, s, j, p) for j, p in zip(jobs, positions))
        return positions

    positions = tuple(job[2][...] for job in jobs)
    positions = lax.fori_loop(0, TICK_ITERS, body, positions)
    for job, pos in zip(jobs, positions):
        job[2][...] = pos


def all_gather_kernel(x_ref, *refs):
    outs = refs[: len(VMEM_TICKS) + 1]
    (
        in_s, in_k, loc_s, loc_k, dec_y, dec_x,
        msg_s, msg_y, msg_x, hdr_s, hdr_y, hdr_x,
        enc_state, dec_stream, dec_pos, counter,
        in_s_sem, in_k_sem, loc_s_sem, loc_k_sem, dec_y_sem, dec_x_sem,
        y_sent, y_landed, x_sent, x_landed, y_credit, x_credit,
    ) = refs[len(outs) :]

    my_x, my_y = lax.axis_index("x"), lax.axis_index("y")
    y_peer, x_peer = (my_x, 1 - my_y), (1 - my_x, my_y)
    send_at = my_x * N_TICKS
    keep_at = (1 - my_x) * N_TICKS
    own_at = my_y * 2 * N_TICKS
    other_at = (1 - my_y) * 2 * N_TICKS

    def load(buf, sem, at, tick):
        slot = tick % N_IN
        rows = pl.ds(pl.multiple_of((at + tick) * TICK_ROWS, TICK_ROWS), TICK_ROWS)
        return pltpu.make_async_copy(x_ref.at[rows], buf.at[slot], sem.at[slot])

    def load_ahead(buf, sem, at, tick):
        @pl.when(tick + N_IN < N_TICKS)
        def _():
            load(buf, sem, at, tick + N_IN).start()

    def store(buf, sem, at, tick):
        slot = tick % N_OUT
        at = at + tick
        for out in outs:

            @pl.when((at >= 0) & (at < out.shape[0]))
            def _(out=out, at=at):
                pltpu.make_async_copy(buf.at[slot], out.at[at], sem.at[slot]).start()

            at = at - out.shape[0]

    def wait_stored(buf, sem, tick):
        slot = tick % N_OUT
        pltpu.make_async_copy(buf.at[slot], buf.at[slot], sem.at[slot]).wait()

    def remote_copy(src, dst, peer, chunk, kind, part):
        (src_hdr, src_msg, sent), (dst_hdr, dst_msg, landed) = src, dst
        i, j = chunk % src_msg.shape[0], chunk % dst_msg.shape[0]
        if kind == HEADER:
            a, b = src_hdr.at[i], dst_hdr.at[j]
        else:
            vregs = {
                PLANES: pl.ds(part * (PLANE_VREGS // 2), PLANE_VREGS // 2),
                STREAMS: pl.ds(STREAM_AT, DENSE_WORDS + 1),
                BINADES: pl.ds(BINADES_AT + part * BINADE_VREGS, BINADE_VREGS),
            }[kind]
            a, b = src_msg.at[i, vregs], dst_msg.at[j, vregs]
        sent_sem = sent.at[i, min(kind, STREAMS)]
        landed_sem = landed.at[j, FIRST_LANDED_SEM[kind] + part]
        return pltpu.make_async_remote_copy(
            a, b, sent_sem, landed_sem, device_id=peer, device_id_type=MESH
        )

    def over_y(chunk, kind, part=0):
        src, dst = (hdr_s, msg_s, y_sent), (hdr_y, msg_y, y_landed)
        return remote_copy(src, dst, y_peer, chunk, kind, part)

    def over_x(chunk, kind, part=0):
        src, dst = (hdr_y, msg_y, x_sent), (hdr_x, msg_x, x_landed)
        return remote_copy(src, dst, x_peer, chunk, kind, part)

    def with_tail(raw, action):
        pl.when(raw == 0)(lambda: action(STREAMS, 0))

        @pl.when(raw != 0)
        def _():
            for part in range(TICKS):
                action(BINADES, part)

    def wait_sent(link, msg, sent, chunk, raw):
        slot = chunk % msg.shape[0]
        planes = msg.at[slot, pl.ds(0, STREAM_AT)]
        link(chunk, HEADER).wait_send()
        pltpu.make_async_copy(planes, planes, sent.at[slot, PLANES]).wait()
        with_tail(raw, lambda kind, part: link(chunk, kind, part).wait_send())

    def send_own(tick):
        chunk, j = tick // TICKS, tick % TICKS
        slot = chunk % N_SEND

        @pl.when((j == 0) & (chunk >= N_SEND))
        def _():
            wait_sent(over_y, msg_s, y_sent, chunk - N_SEND, hdr_s[slot, 1])

        pl.when(tick >= N_OUT)(lambda: wait_stored(loc_s, loc_s_sem, tick))
        load(in_s, in_s_sem, send_at, tick).wait()

        @pl.when(tick == 0)
        def _():
            for i in range(1, N_IN):
                load(in_s, in_s_sem, send_at, i).start()
            for i in range(N_IN):
                load(in_k, in_k_sem, keep_at, i).start()

        x, msg = in_s.at[tick % N_IN], msg_s.at[slot]

        @pl.when(j == 0)
        def _():
            hdr_s[slot, 0] = encode_begin(x, msg, enc_state)

        encode_rows(x, loc_s.at[tick % N_OUT], msg, enc_state, hdr_s[slot, 0], j)
        pl.when(tick == 0)(lambda: pl.semaphore_wait(barrier, 2))
        pl.when((j == 0) & (chunk >= N_RECV))(
            lambda: pl.semaphore_wait(y_credit.at[chunk % N_RECV], 1)
        )

        @pl.when(j == TICKS - 1)
        def _():
            raw = encode_end(msg, enc_state, counter)
            hdr_s[slot, 1] = raw
            over_y(chunk, HEADER).start()
            with_tail(raw, lambda kind, part: over_y(chunk, kind, part).start())

        over_y(chunk, PLANES, 2 * j).start()
        over_y(chunk, PLANES, 2 * j + 1).start()
        store(loc_s, loc_s_sem, own_at + send_at, tick)
        load_ahead(in_s, in_s_sem, send_at, tick)

    def keep_own(tick):
        pl.when(tick >= N_OUT)(lambda: wait_stored(loc_k, loc_k_sem, tick))
        load(in_k, in_k_sem, keep_at, tick).wait()
        loc_k[tick % N_OUT] = in_k[tick % N_IN].astype(BF16)
        store(loc_k, loc_k_sem, own_at + keep_at, tick)
        load_ahead(in_k, in_k_sem, keep_at, tick)

    def relay(tick, half):
        chunk, j = tick // TICKS, tick % TICKS

        def pass_on(kind, part=0):
            over_y(chunk, kind, part).wait_recv()
            over_x(chunk, kind, part).start()

        if half == 0:
            pl.when((j == 0) & (chunk >= N_RECV))(
                lambda: pl.semaphore_wait(x_credit.at[chunk % N_RECV], 1)
            )

            @pl.when(j == TICKS - 1)
            def _():
                pass_on(HEADER)
                with_tail(hdr_y[chunk % N_RECV, 1], pass_on)

        pass_on(PLANES, 2 * j + half)

    def receive(tick):
        chunk, j = tick // TICKS, tick % TICKS
        slot = chunk % N_RECV

        @pl.when(j == 0)
        def _():
            over_x(chunk, HEADER).wait_recv()
            with_tail(
                hdr_x[slot, 1], lambda kind, part: over_x(chunk, kind, part).wait_recv()
            )
            decode_begin(msg_y.at[slot], dec_stream.at[0], dec_pos.at[0], counter)
            decode_begin(msg_x.at[slot], dec_stream.at[1], dec_pos.at[1], counter)

        over_x(chunk, PLANES, 2 * j).wait_recv()
        over_x(chunk, PLANES, 2 * j + 1).wait_recv()
        pl.when(tick >= N_OUT)(lambda: wait_stored(dec_y, dec_y_sem, tick))
        pl.when(tick >= N_OUT)(lambda: wait_stored(dec_x, dec_x_sem, tick))
        jobs = [
            (
                msg.at[slot],
                dec_stream.at[k],
                dec_pos.at[k],
                out.at[tick % N_OUT],
                hdr[slot, 0],
                hdr[slot, 1],
            )
            for k, (msg, hdr, out) in enumerate(
                ((msg_y, hdr_y, dec_y), (msg_x, hdr_x, dec_x))
            )
        ]
        decode_rows(jobs, j)
        store(dec_y, dec_y_sem, other_at + send_at, tick)
        store(dec_x, dec_x_sem, other_at + keep_at, tick)

        @pl.when(j == TICKS - 1)
        def _():
            wait_sent(over_x, msg_y, x_sent, chunk, hdr_y[slot, 1])

            @pl.when(chunk + N_RECV < N_CHUNKS)
            def _():
                for credit, peer in ((y_credit, y_peer), (x_credit, x_peer)):
                    pl.semaphore_signal(
                        credit.at[slot], inc=1, device_id=peer, device_id_type=MESH
                    )

    barrier = pltpu.get_barrier_semaphore()
    load(in_s, in_s_sem, send_at, 0).start()

    def clear_tails(i, _):
        for msg in (msg_y, msg_x):
            for slot in range(N_RECV):
                msg[slot, i] = jnp.zeros((8, 128), I32)

    lax.fori_loop(STREAM_AT, SLOT_VREGS, clear_tails, None)
    for peer in (y_peer, x_peer):
        pl.semaphore_signal(barrier, inc=1, device_id=peer, device_id_type=MESH)
    row = lax.broadcasted_iota(I32, (128, 256), 0)
    col = lax.broadcasted_iota(I32, (128, 256), 1)
    counter[...] = jnp.where(row < col, 1.0, 0.0).astype(BF16)

    def run_tick(tick, _):
        relaying = (tick >= RELAY_LAG) & (tick < N_TICKS + RELAY_LAG)
        pl.when(tick < N_TICKS)(lambda: send_own(tick))
        pl.when(relaying)(lambda: relay(tick - RELAY_LAG, 0))
        pl.when(tick < N_TICKS)(lambda: keep_own(tick))
        pl.when(tick >= DECODE_LAG)(lambda: receive(tick - DECODE_LAG))
        pl.when(relaying)(lambda: relay(tick - RELAY_LAG, 1))

    lax.fori_loop(0, N_TICKS + DECODE_LAG, run_tick, None)

    for chunk in range(N_CHUNKS - N_SEND, N_CHUNKS):
        wait_sent(over_y, msg_s, y_sent, chunk, hdr_s[chunk % N_SEND, 1])
    for tick in range(N_TICKS - N_OUT, N_TICKS):
        wait_stored(loc_s, loc_s_sem, tick)
        wait_stored(loc_k, loc_k_sem, tick)
        wait_stored(dec_y, dec_y_sem, tick)
        wait_stored(dec_x, dec_x_sem, tick)


def pallas_dist_ag_xy_y_m65536_n1024_kernel(x: jax.Array):
    assert x.shape == (SHARD_ROWS, COLS) and x.dtype == jnp.float32
    dma = pltpu.SemaphoreType.DMA
    slots = (N_SEND, N_RECV, N_RECV)
    *pieces, rest = pl.pallas_call(
        all_gather_kernel,
        out_shape=(
            *[pltpu.VMEM((n, TICK_ROWS, COLS), BF16) for n in VMEM_TICKS],
            jax.ShapeDtypeStruct((HBM_TICKS, TICK_ROWS, COLS), BF16),
        ),
        in_specs=[pl.BlockSpec(memory_space=pl.ANY)],
        out_specs=(
            *[pl.BlockSpec(memory_space=pltpu.VMEM) for _ in VMEM_TICKS],
            pl.BlockSpec(memory_space=pl.ANY),
        ),
        scratch_shapes=[
            *[pltpu.VMEM((N_IN, TICK_ROWS, COLS), jnp.float32)] * 2,
            *[pltpu.VMEM((N_OUT, TICK_ROWS, COLS), BF16)] * 4,
            *[pltpu.VMEM((n, SLOT_VREGS, 8, 128), I32) for n in slots],
            *[pltpu.SMEM((n, 2), I32) for n in slots],
            pltpu.VMEM((5, 8, 128), I32),
            pltpu.VMEM((2, STREAM_WORDS, 8, 128), I32),
            pltpu.VMEM((2, 8, 128), I32),
            pltpu.VMEM((128, 256), BF16),
            *[dma((N_IN,))] * 2,
            *[dma((N_OUT,))] * 4,
            dma((N_SEND, 3)),
            dma((N_RECV, 1 + 3 * TICKS)),
            dma((N_RECV, 3)),
            dma((N_RECV, 1 + 3 * TICKS)),
            *[pltpu.SemaphoreType.REGULAR((N_RECV,))] * 2,
        ],
        compiler_params=pltpu.CompilerParams(collective_id=0),
    )(x)

    start = 0
    for n in STAGED_TICKS:
        pieces.append(lax.optimization_barrier(rest[start : start + n]))
        start += n
    return jnp.concatenate([*pieces, rest[start:]]).reshape(2 * SHARD_ROWS, COLS)
```

```python
import jax
import jax.numpy as jnp
import numpy as np
from jax import lax
from jax.experimental import pallas as pl
from jax.experimental.pallas import tpu as pltpu

SHARD_ROWS = 65536
COLS = 1024

TICK_ROWS = 128
TICKS = 4
STREAM_WORDS = 30
DENSE_WORDS = 26
BAND = 8
TOP_OFFSET = 572

RELAY_LAG = 2
DECODE_LAG = 6
N_IN = 2
N_OUT = 2
N_SEND = 2
N_RECV = 3

VMEM_TICKS = (447, 1)
STAGED_TICKS = (281, 293)

CHUNK_ROWS = TICKS * TICK_ROWS
N_TICKS = SHARD_ROWS // 2 // TICK_ROWS
N_CHUNKS = N_TICKS // TICKS
TICK_ITERS = TICK_ROWS // 32
CHUNK_ITERS = TICKS * TICK_ITERS
HBM_TICKS = 4 * N_TICKS - sum(VMEM_TICKS)

HEADER, PLANES, LAST_BITS, STREAMS, BINADES = range(5)
FIRST_LANDED_SEM = (0, 1, 1 + 2 * TICKS, 2 + 2 * TICKS, 1 + 2 * TICKS)

I32 = jnp.int32
BF16 = jnp.bfloat16
MESH = pl.DeviceIdType.MESH
shr = lax.shift_right_logical
shl = lax.shift_left
div, rem = lax.div, lax.rem


def c32(bits):
    return np.uint32(bits & 0xFFFFFFFF).astype(np.int32)


ONES = c32(0x01010101)


def at_least(x, k):
    return shr(x + c32(0x01010101 * (128 - k)), 7) & ONES


def band_base(group):
    typical = shr(group * 209 + 768, 10)
    return lax.clamp(0, typical - BAND // 2, STREAM_WORDS - BAND)


def lane_counts(flags, counter_ref):
    ones = jnp.where(flags, 1.0, 0.0).astype(BF16)
    counts = jnp.dot(ones, counter_ref[...], preferred_element_type=jnp.float32)
    counts = counts.astype(I32)
    return counts[:, :128], counts[:, 128:]


def rows_of(i):
    return pl.ds(pl.multiple_of(i * 32, 32), 32)


def store_word(bits_ref, base, word_idx, word):
    rel = word_idx - base
    pltpu.store(
        bits_ref.at[pl.ds(CHUNK_ITERS + base, BAND)],
        jnp.broadcast_to(word, (BAND, 8, 128)),
        mask=lax.broadcasted_iota(I32, (BAND, 8, 128), 0) == rel,
    )
    return shr(rel, 3)


def encode_begin(x_ref, bits_ref, state_ref):
    w = pltpu.bitcast(x_ref[0:16, :].astype(BF16), I32)
    mean_magnitude = shr(jnp.sum((w & 0x7FFF) + (shr(w, 16) & 0x7FFF)), 14)
    bits_ref[CHUNK_ITERS:] = jnp.zeros((STREAM_WORDS, 8, 128), I32)
    state_ref[...] = jnp.zeros(state_ref.shape, I32)
    return (mean_magnitude + TOP_OFFSET + 0x8000) * 0x10001


def encode_rows(x_ref, loc_ref, message, state_ref, bias, tick):
    planes_ref, bits_ref, binades_ref = message
    top = jnp.full((8, COLS), c32(0x80000000), I32)

    def body(i, carry):
        acc, off, word_idx, bad = carry
        t = tick * TICK_ITERS + i
        b = x_ref[rows_of(i), :].astype(BF16)
        loc_ref[rows_of(i), :] = b
        w = bias - pltpu.bitcast(b, I32)
        ta, tb = w[:8], w[8:]
        planes_ref[t] = (
            (ta & c32(0x007F007F))
            | (shr(ta, 8) & c32(0x00800080))
            | (shl(tb, 8) & c32(0x7F007F00))
            | (tb & c32(0x80008000))
        )
        d = (shr(ta, 7) & c32(0x00FF00FF)) | (shl(tb, 1) & c32(0xFF00FF00))
        binades_ref[t] = d
        ge5 = at_least(d, 5)
        n = (d ^ ((ge5 ^ ONES) * 7)) + ge5 + at_least(d, 11) * 2
        n = n + c32(0x03030303) - at_least(d, 2) * 6
        odd = n & ONES
        p = ((shr(n, 1) & c32(0x1F1F1F1F)) + c32(0x01010100)) * ONES
        last = shr(p, 24)
        unfit = (d & c32(0xC0C0C0C0)) | shr(last, 5)
        last = last & 31
        codes = (
            shr(top, p & 31)
            | shr(top, shr(p, 8) & 31)
            | shr(top, shr(p, 16) & 31)
            | shr(top, last)
        )
        lengths, doubled = last + 1, shl(codes, 1)
        last_bits = 0
        for g in range(8):
            lanes = slice(128 * g, 128 * (g + 1))
            last_bits = last_bits * 2 | odd[:, lanes]
            word = acc | shr(codes[:, lanes], off)
            lost = store_word(bits_ref, band_base(8 * t + g), word_idx, word)
            bad = bad | lost | unfit[:, lanes]
            end = off + lengths[:, lanes]
            full = shr(end, 5)
            acc = lax.select(full != 0, shl(doubled[:, lanes], 31 - off), word)
            off = end & 31
            word_idx = word_idx + full
        bits_ref[t] = last_bits
        return acc, off, word_idx, bad

    state = tuple(state_ref[i] for i in range(state_ref.shape[0]))
    state = lax.fori_loop(0, TICK_ITERS, body, state)
    for i, value in enumerate(state):
        state_ref[i] = value


def encode_end(bits_ref, state_ref, counter_ref):
    acc, off, word_idx, bad = (state_ref[i] for i in range(4))
    lost = store_word(bits_ref, STREAM_WORDS - BAND, word_idx, acc)
    bad = bad | jnp.where(off != 0, lost, 0)

    n_words = word_idx + jnp.where(off != 0, 1, 0)
    pooled = range(DENSE_WORDS, STREAM_WORDS)
    used = jnp.concatenate([n_words > i for i in pooled], axis=0)
    before, total = lane_counts(used, counter_ref)
    lane = lax.broadcasted_iota(I32, used.shape, 1)
    val = jnp.concatenate([bits_ref[CHUNK_ITERS + i] for i in pooled], axis=0)
    move = jnp.where(used, lane - before, 0)
    for k in (1, 2, 4, 8, 16, 32, 64):
        val_in, move_in = pltpu.roll(val, 128 - k, 1), pltpu.roll(move, 128 - k, 1)
        take = (move_in & k) != 0
        val = jnp.where(take, val_in, val)
        move = jnp.where(take, move_in, jnp.where((move & k) != 0, 0, move))
    pool, filled = val[0:8], total[0:8]
    for i in range(1, len(pooled)):
        slot = lane[0:8] - filled
        more = jnp.take_along_axis(val[8 * i : 8 * i + 8], slot & 127, axis=1)
        pool = jnp.where(slot < 0, pool, more)
        filled = filled + total[8 * i : 8 * i + 8]
    bits_ref[CHUNK_ITERS + DENSE_WORDS] = pool
    bad = bad | jnp.where(filled > 128, 1, 0)
    return jnp.max(jnp.where(bad != 0, 1, 0))


def decode_begin(bits_refs, stream_ref, pos_ref, counter_ref):
    dense = pl.ds(CHUNK_ITERS, DENSE_WORDS)
    words = jnp.concatenate([ref[dense] for ref in bits_refs], axis=1)
    stream_ref[:DENSE_WORDS] = words
    seen = jnp.sum(lax.population_count(words), axis=0)
    pool = jnp.concatenate([ref[CHUNK_ITERS + DENSE_WORDS] for ref in bits_refs])
    filled = 0
    for i in range(DENSE_WORDS, STREAM_WORDS):
        used = seen < CHUNK_ROWS
        before, total = lane_counts(used, counter_ref)
        word = jnp.take_along_axis(pool, (filled + before) & 127, axis=1)
        word = jnp.where(used, word, 0)
        stream_ref[i] = word
        seen = seen + lax.population_count(word)
        filled = filled + total
    stream_ref[STREAM_WORDS:] = jnp.zeros((2, *pos_ref.shape), I32)
    pos_ref[...] = jnp.zeros(pos_ref.shape, I32)


def decode_rows(messages, headers, out_refs, stream_ref, pos_ref, tick):
    top = jnp.full(pos_ref.shape, c32(0x80000000), I32)

    def body(i, pos):
        t = tick * TICK_ITERS + i
        ones_at = []
        for g in range(0, 8, 2):
            base = band_base(8 * t + g)
            rel, off = shr(pos, 5) - base, pos & 31
            near = stream_ref[pl.ds(base, BAND + 2)]
            for bit in (4, 2, 1):
                near = jnp.where((rel & bit) != 0, near[bit:], near[:-bit])
            window = shl(near[:2], off[None]) | shr(shr(near[1:], 1), 31 - off[None])
            bits = window[0]
            for h in range(2):
                p0 = lax.clz(bits)
                rest = bits ^ shr(top, p0)
                p1 = lax.clz(rest)
                rest = rest ^ shr(top, p1)
                p2 = lax.clz(rest)
                rest = rest ^ shr(top, p2)
                p3 = lax.clz(rest)
                if h == 0:
                    bits = shl(shl(bits, 1), p3) | shr(window[1], 31 - p3)
                pos = pos + p3 + 1
                ones_at.append(p0 | shl(p1, 8) | shl(p2, 16) | shl(p3, 24))
        twice = jnp.concatenate(ones_at, axis=1) * c32(2 - 512) - c32(0x02020200)
        for k, (planes_ref, bits_ref, binades_ref) in enumerate(messages):
            bias, raw = headers[k]
            last_bits = bits_ref[t]
            odd = jnp.concatenate([shr(last_bits, 7 - g) for g in range(8)], axis=1)
            n = twice[8 * k : 8 * k + 8] | (odd & ONES)
            ge3, ge9, ge11 = at_least(n, 3), at_least(n, 9), at_least(n, 11)
            d = (n ^ ((ge3 ^ ge9 ^ ge11 ^ ONES) * 3)) + ge3 + ONES
            d = d + ge11 * 9 - ge9 * 11
            d = jnp.where(raw != 0, binades_ref[t], d)
            low = planes_ref[t]
            ta = (
                (low & c32(0x007F007F))
                | (shl(low, 8) & c32(0x80008000))
                | (shl(d, 7) & c32(0x7F807F80))
            )
            tb = (
                (shr(low, 8) & c32(0x007F007F))
                | (low & c32(0x80008000))
                | (shr(d, 1) & c32(0x7F807F80))
            )
            w = bias - jnp.concatenate([ta, tb])
            out_refs[k][rows_of(i), :] = pltpu.bitcast(w, BF16)
        return pos

    pos_ref[...] = lax.fori_loop(0, TICK_ITERS, body, pos_ref[...])


def all_gather_kernel(x_ref, *refs):
    outs = refs[: len(VMEM_TICKS) + 1]
    (
        in_s, in_k, loc_s, loc_k, dec_y, dec_x,
        msg_s, msg_y, msg_x, hdr_s, hdr_y, hdr_x,
        enc_state, dec_stream, dec_pos, counter,
        in_s_sem, in_k_sem, loc_s_sem, loc_k_sem, dec_y_sem, dec_x_sem,
        y_sent, y_landed, x_sent, x_landed, y_credit, x_credit,
    ) = refs[len(outs) :]

    my_x, my_y = lax.axis_index("x"), lax.axis_index("y")
    y_peer, x_peer = (my_x, 1 - my_y), (1 - my_x, my_y)
    send_at = my_x * N_TICKS
    keep_at = (1 - my_x) * N_TICKS
    own_at = my_y * 2 * N_TICKS
    other_at = (1 - my_y) * 2 * N_TICKS

    def load(buf, sem, at, tick):
        slot = rem(tick, N_IN)
        rows = pl.ds(pl.multiple_of((at + tick) * TICK_ROWS, TICK_ROWS), TICK_ROWS)
        return pltpu.make_async_copy(x_ref.at[rows], buf.at[slot], sem.at[slot])

    def load_ahead(buf, sem, at, tick):
        @pl.when(tick + N_IN < N_TICKS)
        def _():
            load(buf, sem, at, tick + N_IN).start()

    def store(buf, sem, at, tick):
        slot = rem(tick, N_OUT)
        at = at + tick
        for out in outs:

            @pl.when((at >= 0) & (at < out.shape[0]))
            def _(out=out, at=at):
                pltpu.make_async_copy(buf.at[slot], out.at[at], sem.at[slot]).start()

            at = at - out.shape[0]

    def wait_stored(buf, sem, tick):
        slot = rem(tick, N_OUT)
        pltpu.make_async_copy(buf.at[slot], buf.at[slot], sem.at[slot]).wait()

    def remote_copy(src, dst, peer, chunk, kind, part):
        (src_hdr, src_msg, sent), (dst_hdr, dst_msg, landed) = src, dst
        i, j = rem(chunk, src_hdr.shape[0]), rem(chunk, dst_hdr.shape[0])
        if kind == HEADER:
            a, b = src_hdr.at[i], dst_hdr.at[j]
        else:
            k, at = {
                PLANES: (0, pl.ds(part * (TICK_ITERS // 2), TICK_ITERS // 2)),
                LAST_BITS: (1, pl.ds(0, CHUNK_ITERS)),
                STREAMS: (1, pl.ds(CHUNK_ITERS, DENSE_WORDS + 1)),
                BINADES: (2, pl.ds(part * TICK_ITERS, TICK_ITERS)),
            }[kind]
            a, b = src_msg[k].at[i, at], dst_msg[k].at[j, at]
        sent_sem = sent.at[i, min(kind, LAST_BITS)]
        landed_sem = landed.at[j, FIRST_LANDED_SEM[kind] + part]
        return pltpu.make_async_remote_copy(
            a, b, sent_sem, landed_sem, device_id=peer, device_id_type=MESH
        )

    def over_y(chunk, kind, part=0):
        src, dst = (hdr_s, msg_s, y_sent), (hdr_y, msg_y, y_landed)
        return remote_copy(src, dst, y_peer, chunk, kind, part)

    def over_x(chunk, kind, part=0):
        src, dst = (hdr_y, msg_y, x_sent), (hdr_x, msg_x, x_landed)
        return remote_copy(src, dst, x_peer, chunk, kind, part)

    def with_tail(raw, action):
        @pl.when(raw == 0)
        def _():
            action(STREAMS, 0)
            action(LAST_BITS, 0)

        @pl.when(raw != 0)
        def _():
            for part in range(TICKS):
                action(BINADES, part)

    def wait_sent(link, chunk, raw):
        link(chunk, HEADER).wait_send()
        for part in range(2 * TICKS):
            link(chunk, PLANES, part).wait_send()
        with_tail(raw, lambda kind, part: link(chunk, kind, part).wait_send())

    def send_own(tick):
        chunk, j = div(tick, TICKS), rem(tick, TICKS)
        slot = rem(chunk, N_SEND)

        @pl.when((j == 0) & (chunk >= N_SEND))
        def _():
            wait_sent(over_y, chunk - N_SEND, hdr_s[slot, 1])

        pl.when(tick >= N_OUT)(lambda: wait_stored(loc_s, loc_s_sem, tick))
        load(in_s, in_s_sem, send_at, tick).wait()

        @pl.when(tick == 0)
        def _():
            for i in range(1, N_IN):
                load(in_s, in_s_sem, send_at, i).start()
            for i in range(N_IN):
                load(in_k, in_k_sem, keep_at, i).start()

        x, msg = in_s.at[rem(tick, N_IN)], [m.at[slot] for m in msg_s]

        @pl.when(j == 0)
        def _():
            hdr_s[slot, 0] = encode_begin(x, msg[1], enc_state)

        encode_rows(x, loc_s.at[rem(tick, N_OUT)], msg, enc_state, hdr_s[slot, 0], j)
        pl.when(tick == 0)(lambda: pl.semaphore_wait(barrier, 2))
        pl.when((j == 0) & (chunk >= N_RECV))(
            lambda: pl.semaphore_wait(y_credit.at[rem(chunk, N_RECV)], 1)
        )

        @pl.when(j == TICKS - 1)
        def _():
            raw = encode_end(msg[1], enc_state, counter)
            hdr_s[slot, 1] = raw
            over_y(chunk, HEADER).start()
            with_tail(raw, lambda kind, part: over_y(chunk, kind, part).start())

        over_y(chunk, PLANES, 2 * j).start()
        over_y(chunk, PLANES, 2 * j + 1).start()
        store(loc_s, loc_s_sem, own_at + send_at, tick)
        load_ahead(in_s, in_s_sem, send_at, tick)

    def keep_own(tick):
        pl.when(tick >= N_OUT)(lambda: wait_stored(loc_k, loc_k_sem, tick))
        load(in_k, in_k_sem, keep_at, tick).wait()
        loc_k[rem(tick, N_OUT)] = in_k[rem(tick, N_IN)].astype(BF16)
        store(loc_k, loc_k_sem, own_at + keep_at, tick)
        load_ahead(in_k, in_k_sem, keep_at, tick)

    def relay(tick, half):
        chunk, j = div(tick, TICKS), rem(tick, TICKS)

        def pass_on(kind, part=0):
            over_y(chunk, kind, part).wait_recv()
            over_x(chunk, kind, part).start()

        if half == 0:
            pl.when((j == 0) & (chunk >= N_RECV))(
                lambda: pl.semaphore_wait(x_credit.at[rem(chunk, N_RECV)], 1)
            )

            @pl.when(j == TICKS - 1)
            def _():
                pass_on(HEADER)
                with_tail(hdr_y[rem(chunk, N_RECV), 1], pass_on)

        pass_on(PLANES, 2 * j + half)

    def receive(tick):
        chunk, j = div(tick, TICKS), rem(tick, TICKS)
        slot = rem(chunk, N_RECV)

        @pl.when(j == 0)
        def _():
            over_x(chunk, HEADER).wait_recv()
            raw = hdr_x[slot, 1]
            pl.when(raw == 0)(lambda: over_x(chunk, STREAMS).wait_recv())
            bits = [msg[1].at[slot] for msg in (msg_y, msg_x)]
            decode_begin(bits, dec_stream, dec_pos, counter)
            pl.when(raw == 0)(lambda: over_x(chunk, LAST_BITS).wait_recv())

            @pl.when(raw != 0)
            def _():
                for part in range(TICKS):
                    over_x(chunk, BINADES, part).wait_recv()

        over_x(chunk, PLANES, 2 * j).wait_recv()
        over_x(chunk, PLANES, 2 * j + 1).wait_recv()
        pl.when(tick >= N_OUT)(lambda: wait_stored(dec_y, dec_y_sem, tick))
        pl.when(tick >= N_OUT)(lambda: wait_stored(dec_x, dec_x_sem, tick))
        decode_rows(
            [[m.at[slot] for m in msg] for msg in (msg_y, msg_x)],
            [(hdr[slot, 0], hdr[slot, 1]) for hdr in (hdr_y, hdr_x)],
            [out.at[rem(tick, N_OUT)] for out in (dec_y, dec_x)],
            dec_stream,
            dec_pos,
            j,
        )
        store(dec_y, dec_y_sem, other_at + send_at, tick)
        store(dec_x, dec_x_sem, other_at + keep_at, tick)

        @pl.when(j == TICKS - 1)
        def _():
            wait_sent(over_x, chunk, hdr_y[slot, 1])

            @pl.when(chunk + N_RECV < N_CHUNKS)
            def _():
                for credit, peer in ((y_credit, y_peer), (x_credit, x_peer)):
                    pl.semaphore_signal(
                        credit.at[slot], inc=1, device_id=peer, device_id_type=MESH
                    )

    barrier = pltpu.get_barrier_semaphore()
    load(in_s, in_s_sem, send_at, 0).start()

    for _, bits, binades in (msg_y, msg_x):
        bits[...] = jnp.zeros(bits.shape, I32)
        binades[...] = jnp.zeros(binades.shape, I32)
    for peer in (y_peer, x_peer):
        pl.semaphore_signal(barrier, inc=1, device_id=peer, device_id_type=MESH)
    row = lax.broadcasted_iota(I32, (128, 256), 0)
    col = lax.broadcasted_iota(I32, (128, 256), 1)
    counter[...] = jnp.where(row < col, 1.0, 0.0).astype(BF16)

    def run_tick(tick, _):
        relaying = (tick >= RELAY_LAG) & (tick < N_TICKS + RELAY_LAG)
        pl.when(tick < N_TICKS)(lambda: send_own(tick))
        pl.when(relaying)(lambda: relay(tick - RELAY_LAG, 0))
        pl.when(tick < N_TICKS)(lambda: keep_own(tick))
        pl.when(tick >= DECODE_LAG)(lambda: receive(tick - DECODE_LAG))
        pl.when(relaying)(lambda: relay(tick - RELAY_LAG, 1))

    lax.fori_loop(0, N_TICKS + DECODE_LAG, run_tick, None)

    for chunk in range(N_CHUNKS - N_SEND, N_CHUNKS):
        wait_sent(over_y, chunk, hdr_s[chunk % N_SEND, 1])
    for tick in range(N_TICKS - N_OUT, N_TICKS):
        wait_stored(loc_s, loc_s_sem, tick)
        wait_stored(loc_k, loc_k_sem, tick)
        wait_stored(dec_y, dec_y_sem, tick)
        wait_stored(dec_x, dec_x_sem, tick)


def pallas_dist_ag_xy_y_m65536_n1024_kernel(x: jax.Array):
    assert x.shape == (SHARD_ROWS, COLS) and x.dtype == jnp.float32
    dma = pltpu.SemaphoreType.DMA
    slots = (N_SEND, N_RECV, N_RECV)
    *pieces, rest = pl.pallas_call(
        all_gather_kernel,
        out_shape=(
            *[pltpu.VMEM((n, TICK_ROWS, COLS), BF16) for n in VMEM_TICKS],
            jax.ShapeDtypeStruct((HBM_TICKS, TICK_ROWS, COLS), BF16),
        ),
        in_specs=[pl.BlockSpec(memory_space=pl.ANY)],
        out_specs=(
            *[pl.BlockSpec(memory_space=pltpu.VMEM) for _ in VMEM_TICKS],
            pl.BlockSpec(memory_space=pl.ANY),
        ),
        scratch_shapes=[
            *[pltpu.VMEM((N_IN, TICK_ROWS, COLS), jnp.float32)] * 2,
            *[pltpu.VMEM((N_OUT, TICK_ROWS, COLS), BF16)] * 4,
            *[
                (
                    pltpu.VMEM((n, CHUNK_ITERS, 8, COLS), I32),
                    pltpu.VMEM((n, CHUNK_ITERS + STREAM_WORDS, 8, 128), I32),
                    pltpu.VMEM((n, CHUNK_ITERS, 8, COLS), I32),
                )
                for n in slots
            ],
            *[pltpu.SMEM((n, 2), I32) for n in slots],
            pltpu.VMEM((4, 8, 128), I32),
            pltpu.VMEM((STREAM_WORDS + 2, 16, 128), I32),
            pltpu.VMEM((16, 128), I32),
            pltpu.VMEM((128, 256), BF16),
            *[dma((N_IN,))] * 2,
            *[dma((N_OUT,))] * 4,
            dma((N_SEND, 3)),
            dma((N_RECV, 1 + 3 * TICKS)),
            dma((N_RECV, 3)),
            dma((N_RECV, 1 + 3 * TICKS)),
            *[pltpu.SemaphoreType.REGULAR((N_RECV,))] * 2,
        ],
        compiler_params=pltpu.CompilerParams(collective_id=0),
    )(x)

    start = 0
    for n in STAGED_TICKS:
        pieces.append(lax.optimization_barrier(rest[start : start + n]))
        start += n
    return jnp.concatenate([*pieces, rest[start:]]).reshape(2 * SHARD_ROWS, COLS)
```
